```python
import numpy as np

kernel_name = "dist_sparse_attn_localglobal_htp_kvseq_b2_sq256_skv256_hq4_dh64"

def setup_inputs():
    x = np.random.randn(2, 256, 512).astype(np.float32)
    Wq = np.random.randn(512, 1024).astype(np.float32) * 0.02
    K_ext = np.random.randn(2, 1024, 16, 64).astype(np.float32)
    V_ext = np.random.randn(2, 1024, 16, 64).astype(np.float32)
    Wo = np.random.randn(1024, 512).astype(np.float32) * 0.02
    return {"x": x, "Wq": Wq, "K_ext": K_ext, "V_ext": V_ext, "Wo": Wo}

def reference(x, Wq, K_ext, V_ext, Wo):
    B, Sq, Skv, Hq, Dh = 2, 256, 1024, 16, 64
    Q = (x @ Wq).reshape(B, Sq, Hq, Dh)
    qi = np.arange(Sq)[:, None]
    ki = np.arange(Skv)[None, :]
    local = np.abs(qi - ki) <= 128
    glob = (ki < 32) | (qi < 32)
    mask = local | glob
    scores = np.einsum('bihd,bjhd->bhij', Q, K_ext).astype(np.float32) * 0.125
    scores = np.where(mask[None, None, :, :], scores, -1e9)
    scores_max = scores.max(axis=-1, keepdims=True)
    w = np.exp(scores - scores_max)
    row_keep = mask.any(axis=1)
    w_sum = np.where(row_keep[None, None, :, None], w.sum(axis=-1, keepdims=True), 1.0)
    w = w / w_sum
    w = np.where(row_keep[None, None, :, None], w, 0.0)
    ctx = np.einsum('bhij,bjhd->bihd', w, V_ext).reshape(B, Sq, Hq * Dh)
    return ctx @ Wo
```

```python
import re

import jax
import jax.numpy as jnp
from jax import lax
from jax.experimental import pallas as pl
from jax.experimental.pallas import tpu as pltpu

F32 = jnp.float32
BF16 = jnp.bfloat16
MESH = pl.DeviceIdType.MESH
LOG2E = 1.4426950408889634
QSCALE = 0.125 * LOG2E
NEG = -1e9 * LOG2E
TI = {"H0": 0, "H1": 1, "L0": 2, "L1": 3}
PVR = 32
ATT = ("att0", "att1", "att01", "gatt")


def _parts(it):
    if it.startswith("cq"):
        return ("h",)
    if it.startswith(("c0_", "c1_")):
        return ("t", "l2")
    if it.startswith(("gp", "gacc")):
        return ("h", "l1")
    if it.startswith(("q", "m_")) or re.match(r"[kvw]\d_", it):
        return ("t",)
    if it[0] in "PS":
        return ("ar",)
    return ()


def make_kernel(PROG, NCH, SPLIT):
    CW = 512 * 8 // NCH

    def chunk(k):
        r, o = divmod(k * CW, 512)
        return r * 16, o

    POOLS = ("t", "h", "l2", "l1", "ar")
    slots = {c: {k: {} for k in POOLS} for c in range(4)}

    def slot(c, it):
        for k in _parts(it):
            slots[c][k].setdefault(it, len(slots[c][k]))

    nrecv = [0] * 4
    nsent = {c: {k: 0 for k in POOLS} for c in range(4)}
    recv_of = {c: {} for c in range(4)}
    for c in range(4):
        for st in PROG[c]:
            for op in st:
                if op[0] == "s":
                    _, it, d, dit = op
                    n = len(_parts(it))
                    recv_of[d][dit] = list(range(nrecv[d], nrecv[d] + n))
                    nrecv[d] += n
                    for k in _parts(it):
                        nsent[c][k] += 1
                    slot(d, dit)
                    slot(c, it)
                elif op[0] == "c" and not op[1].startswith(("zmerge", "pfin", "add")):
                    for it in op[3]:
                        slot(c, it)
    nsl = {k: max(1, max(max(len(slots[c][k]), nsent[c][k]) for c in range(4))) for k in POOLS}
    nload = max(sum(op[0] == "l" for st in PROG[c] for op in st) for c in range(4))

    def body(x_hbm, wq_hbm, k_hbm, v_hbm, wo_hbm, out_ref,
             xr, wqr, kr, vr, wor, wo, pacc, tb, hb, l2b, l1b, arb,
             ssem, rsem, lsem, rdy, mark):
        me = lax.axis_index("i")
        bar = pltpu.get_barrier_semaphore()
        pool = dict(zip(POOLS, (tb, hb, l2b, l1b, arb)))

        def lanes(rows):
            return lax.broadcasted_iota(jnp.int32, (rows, 128), 1)

        def rows_of(t):
            return int(t[1]), (128 if t[0] == "H" else 0)

        def load_parts(name):
            w = name.split("_")
            if w[1] == "x":
                b, r = rows_of(w[2])
                return [(x_hbm.at[b, pl.ds(r, 128), :], xr.at[b, pl.ds(r, 128), :])]
            if w[1] == "wq":
                o = 128 * "ab".index(w[2][0])
                rows = pl.ds(128 * int(w[2][1]), 128) if len(w[2]) > 1 else pl.ds(0, 512)
                return [(wq_hbm.at[rows, pl.ds(o, 128)], wqr.at[rows, pl.ds(o, 128)])]
            if w[1] == "wo":
                o = 128 * "ab".index(w[2][0]) + 64 * int(w[2][1])
                return [(wo_hbm.at[pl.ds(o, 64), :], wor.at[pl.ds(o, 64), :])]
            g, pr, b = int(w[2][0]), "ab".index(w[2][1]), int(w[2][2])
            o = g * 256 + pr * 128
            srcs = {"k": (k_hbm, kr), "v": (v_hbm, vr)}
            return [(srcs[a][0].at[b, pl.ds(o, 128), :], srcs[a][1].at[b, pl.ds(o, 128), :]) for a in w[1]]

        def refs_of(c, it):
            return [pool[k].at[slots[c][k][it]] for k in _parts(it)]

        def program(c):
            waited, known, staged, consumed = set(), set(), set(), set()
            ldesc, vals, lazy, pstate = {}, {}, {}, {}
            sent_items = {op[1] for st in PROG[c] for op in st if op[0] == "s"}
            nl = [0]

            def ref(it):
                return refs_of(c, it)[0]

            def sig(sem, d):
                pl.semaphore_signal(sem, inc=1, device_id=(d,), device_id_type=MESH)

            def load_descs(name):
                return [pltpu.make_async_copy(src, dst, lsem.at[ldesc[name] + i])
                        for i, (src, dst) in enumerate(load_parts(name))]

            def start_loads(names):
                for name in names:
                    ldesc[name] = nl[0]
                    for cp in load_descs(name):
                        nl[0] += 1
                        cp.start()

            def prologue():
                first = [op[1] for op in PROG[c][0]]
                if c == 0:
                    sig(bar, 1)
                    sig(bar, 3)
                    start_loads(first)
                elif c in (1, 3):
                    sig(bar, 0)
                    start_loads(first[:2])
                    pl.semaphore_wait(bar, 1)
                    sig(bar, 2)
                    known.add(0)
                    start_loads(first[2:])
                else:
                    start_loads(first[:2])
                    pl.semaphore_wait(bar, 2)
                    known.update((0, 1, 3))
                    for d in (1, 3, 0):
                        sig(rdy, d)
                    start_loads(first[2:])

            def need_peer(d):
                if d in known:
                    return
                if c == 0 and 1 not in known:
                    pl.semaphore_wait(bar, 2)
                    known.update((1, 3))
                if d not in known:
                    pl.semaphore_wait(rdy, 1)
                    known.update((0, 1, 2, 3))

            def wait_item(it):
                if it in waited:
                    return
                waited.add(it)
                if it in ldesc:
                    for cp in load_descs(it):
                        cp.wait()
                elif it in recv_of[c]:
                    for r, ri in zip(refs_of(c, it), recv_of[c][it]):
                        pltpu.make_async_remote_copy(
                            src_ref=r, dst_ref=r, send_sem=ssem.at[0], recv_sem=rsem.at[ri],
                            device_id=(c,), device_id_type=MESH).wait_recv()

            def do_send(it, d, dit):
                for k, rs, rd, ri in zip(_parts(it), refs_of(c, it), refs_of(d, dit), recv_of[d][dit]):
                    pltpu.make_async_remote_copy(
                        src_ref=rs, dst_ref=rd, send_sem=ssem.at[POOLS.index(k)], recv_sem=rsem.at[ri],
                        device_id=(d,), device_id_type=MESH).start()

            def kv_tiles(ins, a, n=None):
                out = []
                for it in ins:
                    if it.startswith("raw_" + a):
                        key = it.split("_")[2]
                        o, b = int(key[0]) * 256 + 128 * "ab".index(key[1]), int(key[2])
                        src = kr if a == "k" else vr
                        for h in range(n or 2):
                            out.append(lambda r0, r1, o=o, b=b, h=h, src=src:
                                       src[b, o + r0:o + r1, h * 128:(h + 1) * 128].astype(BF16))
                    elif it[0] == a and it[1].isdigit():
                        out.append(lambda r0, r1, it=it: ref(it)[r0:r1, :])
                return out

            def tdot(a, b):
                return lax.dot_general(a, b, (((0,), (0,)), ((), ())), preferred_element_type=F32)

            def att_a(name, ins):
                typ, key = name.split()
                ki = lax.broadcasted_iota(jnp.int32, (128, 128), 0)
                qi = lax.broadcasted_iota(jnp.int32, (128, 128), 1)
                n = 1 if c == 1 else 2
                ks = [it for it in ins[1:] if it[0] == "k"]
                vs = kv_tiles(ins[1:], "v", n)
                z = jnp.zeros((64, 128), BF16)
                res = []
                for j in range(2):
                    q = ref(ins[0])[j * 64:(j + 1) * 64, :]
                    w = jnp.concatenate([q, z] if j == 0 else [z, q], axis=0)
                    blocks = [jnp.concatenate([jnp.dot(ref(it)[r:r + 64, :], w, preferred_element_type=F32)
                                               for r in (0, 64)], axis=0) for it in ks]
                    if typ != "att1":
                        if key[2] == "L":
                            blocks[1] = jnp.where((ki <= qi) | (qi < 32), blocks[1], NEG)
                        else:
                            blocks[0] = jnp.where((ki >= qi) | (ki < 32), blocks[0], NEG)
                    if typ != "att0":
                        blocks[-1] = jnp.where(ki <= qi, blocks[-1], NEG)
                    s = jnp.concatenate(blocks, axis=0)
                    res.append((s, jnp.max(s, axis=0, keepdims=True)))
                return res, vs

            def att_b(res, vs, out):
                r = refs_of(c, out)
                lses = []
                for j, (s, m) in enumerate(res):
                    p = jnp.exp2(s - m)
                    l = jnp.sum(p, axis=0, keepdims=True)
                    pb = p.astype(BF16)
                    inv = 1.0 / l
                    for o in range(j * 64, (j + 1) * 64, PVR):
                        vt = jnp.concatenate([v(o, o + PVR) for v in vs], axis=1)
                        r[0][o:o + PVR, :] = (jnp.dot(vt, pb, preferred_element_type=F32) * inv).astype(BF16)
                    lses.append(m + jnp.log2(l))
                r[1][...] = jnp.concatenate(lses, axis=0)

            def gatt_a(name, ins):
                cqv = ref(ins[0])[...]
                lane = lanes(64)
                z = jnp.zeros_like(cqv)
                ws = [jnp.where((lane >= 32 * h) & (lane < 32 * h + 32), cqv, z) for h in range(4)]
                wa, wb = jnp.concatenate(ws[:2], axis=0), jnp.concatenate(ws[2:], axis=0)
                ks, vs = kv_tiles(ins[1:], "k"), kv_tiles(ins[1:], "v")
                s = jnp.concatenate([tdot(ks[h](0, 128), wa) + tdot(ks[2 + h](0, 128), wb) for h in range(2)], axis=0)
                return s, jnp.max(s, axis=0, keepdims=True), vs

            def gatt_b(s, m, vs, out):
                p = jnp.exp2(s - m)
                l = jnp.sum(p, axis=0, keepdims=True)
                pb = p.astype(BF16)
                cs = jnp.concatenate(
                    [jnp.dot(jnp.concatenate([vs[2 * p_](0, 128), vs[2 * p_ + 1](0, 128)], axis=1), pb,
                             preferred_element_type=F32) for p_ in range(2)], axis=0)
                acc = cs[:64]
                for h in range(1, 4):
                    acc = jnp.where(lanes(64) >= 32 * h, cs[h * 64:(h + 1) * 64], acc)
                r = refs_of(c, out)
                r[0][...] = (acc * (1.0 / l)).astype(BF16)
                r[1][...] = m + jnp.log2(l)

            def merge_w(lses):
                mx = lses[0]
                for a in lses[1:]:
                    mx = jnp.maximum(mx, a)
                ws = [jnp.exp2(a - mx) for a in lses]
                tot = ws[0]
                for a in ws[1:]:
                    tot = tot + a
                inv = 1.0 / tot
                return [a * inv for a in ws], mx + jnp.log2(tot)

            def merged_pair(i0, i1):
                r0, r1 = refs_of(c, i0), refs_of(c, i1)
                ws, _ = merge_w([r0[1][...], r1[1][...]])
                outs = []
                for j in range(2):
                    sl = slice(j * 64, (j + 1) * 64)
                    outs.append(r0[0][sl, :].astype(F32) * ws[0][j:j + 1] + r1[0][sl, :].astype(F32) * ws[1][j:j + 1])
                return jnp.concatenate(outs, axis=0)

            def compact(rows, ln):
                acc = rows[0]
                for h in range(1, 4):
                    acc = jnp.where(ln >= 32 * h, pltpu.roll(rows[h], 32 * h, 1), acc)
                return acc

            def ar_val(it):
                if it in vals:
                    return vals[it]
                m_ = re.match(r"P([HL][01])_(\d+)_\d$", it)
                if m_:
                    r, o = chunk(int(m_.group(2)))
                    return pacc[TI[m_.group(1)], r:r + 16, o:o + CW]
                return ref(it)[...].astype(F32)

            def compute(name, ins, outs):
                typ, *w = name.split()
                key = w[0]
                if typ == "cvt":
                    o = 128 * "ab".index(key[2]) + 64 * int(key[3])
                    wo[o:o + 64, :] = wor[o:o + 64, :].astype(BF16)
                elif typ == "cvtq":
                    o, r = 128 * "ab".index(key[1]), 128 * int(key[2])
                    ref(outs[0])[...] = wqr[r:r + 128, o:o + 128].astype(BF16)
                elif typ == "qproj":
                    b, r = rows_of(key[2:4])
                    if len(ins) > 2:
                        wq = jnp.concatenate([ref(it)[...] for it in ins[1:]], axis=0)
                    else:
                        o = 128 * "ab".index(key[1])
                        wq = wqr[:, o:o + 128].astype(BF16)
                    q = lax.dot_general(wq, xr[b, r:r + 128, :].astype(BF16), (((0,), (1,)), ((), ())),
                                        preferred_element_type=F32)
                    ref(outs[0])[...] = (q * QSCALE).astype(BF16)
                elif typ == "cq":
                    rows = [ref(ins[h // 2])[(h % 2) * 64:(h % 2) * 64 + 64, :].astype(F32) for h in range(4)]
                    ref(outs[0])[...] = compact(rows, lanes(64)).astype(BF16)
                elif typ == "vprep":
                    for it, ld in zip(outs, kv_tiles(ins, "v")):
                        ref(it)[...] = ld(0, 128)
                elif typ == "kprep":
                    o, b = int(key[0]) * 256 + 128 * "ab".index(key[1]), int(key[2])
                    for h, it in enumerate(outs):
                        ref(it)[...] = kr[b, o:o + 128, h * 128:(h + 1) * 128].T.astype(BF16)
                elif typ == "merge":
                    ref(outs[0])[...] = merged_pair(*ins).astype(BF16)
                elif typ in ("zmerge", "gfinal"):
                    lazy[outs[0]] = ins
                elif typ == "proj":
                    t = key[2:4]
                    o = 128 * "ab".index(key[1])
                    ct = merged_pair(*lazy[ins[0]]) if ins[0] in lazy else ref(ins[0])[...]
                    r0 = 32 if t[0] == "L" else 0
                    p = tdot(ct.astype(BF16), wo[o:o + 128, :])[r0:]
                    if pstate.get(t):
                        p = p + pacc[TI[t], r0:, :]
                    pstate[t] = True
                    pacc[TI[t], r0:, :] = p
                elif typ == "pfin":
                    pass
                elif typ == "pfing":
                    rs = [refs_of(c, ins[h // 2]) for h in range(4)]
                    lacc = compact([r[1][(h % 2):(h % 2) + 1, :] for h, r in enumerate(rs)], lanes(1))
                    others = [refs_of(c, it) for it in lazy[ins[2]]]
                    ws, _ = merge_w([lacc] + [r[1][...] for r in others])
                    cm = None
                    for r, w_ in zip(others, ws[1:]):
                        a = r[0][...].astype(F32) * w_
                        cm = a if cm is None else cm + a
                    xs = []
                    for h, r in enumerate(rs):
                        back = (lambda a: pltpu.roll(a, 128 - 32 * h, 1)) if h else (lambda a: a)
                        xs.append(r[0][(h % 2) * 64:(h % 2) * 64 + 64, :].astype(F32) * back(ws[0]) + back(cm))
                    xt = jnp.concatenate(xs, axis=0).astype(BF16)
                    pacc[TI[key], 0:32, :] = tdot(xt[:, :32], wo[...])
                elif typ == "gmerge":
                    rs = [refs_of(c, it) for it in ins]
                    ws, lse = merge_w([r[1][...] for r in rs])
                    cm = None
                    for r, w_ in zip(rs, ws):
                        a = r[0][...].astype(F32) * w_
                        cm = a if cm is None else cm + a
                    ro = refs_of(c, outs[0])
                    ro[0][...] = cm.astype(BF16)
                    ro[1][...] = lse
                elif typ == "add":
                    v = ar_val(ins[0])
                    for it in ins[1:]:
                        v = v + ar_val(it)
                    vals[outs[0]] = v
                    if outs[0] in sent_items:
                        ref(outs[0])[...] = v.astype(BF16)
                elif typ == "out":
                    b, r0 = rows_of(key[:2])
                    r, o = chunk(int(key[3:]))
                    out_ref[b, r0 + r:r0 + r + 16, o:o + CW] = ar_val(ins[0])
                    consumed.add(ins[0])
                else:
                    raise ValueError(name)

            def run_step(st):
                start_loads([op[1] for op in st if op[0] == "l"])
                comp = [op for op in st if op[0] == "c"]
                sends = [op for op in st if op[0] == "s"]
                local = {o for op in comp for o in op[3]}
                for op in st:
                    if op[0] == "c":
                        for it in op[2]:
                            if it not in local:
                                wait_item(it)
                    elif op[0] == "s":
                        need_peer(op[2])
                        if op[1] not in local:
                            wait_item(op[1])
                head = [op for op in comp if op[1].split()[0] in ATT and not any(it in local for it in op[2])]
                pend = {}

                def flush():
                    for o, (f, a) in pend.items():
                        f(*a, o)
                    pend.clear()

                for op in head + [op for op in comp if op not in head]:
                    _, name, ins, outs = op
                    if any(it in pend for it in ins):
                        flush()
                    typ = name.split()[0]
                    if typ == "gatt":
                        pend[outs[0]] = (gatt_b, gatt_a(name, ins))
                    elif typ in ATT:
                        pend[outs[0]] = (att_b, att_a(name, ins))
                    else:
                        compute(name, ins, outs)
                flush()
                for op in sends:
                    if op[1][0] == "P" and op[1] not in staged:
                        staged.add(op[1])
                        ref(op[1])[...] = ar_val(op[1]).astype(BF16)
                    do_send(op[1], op[2], op[3])
                for it in list(vals):
                    if it in sent_items or it in consumed:
                        del vals[it]

            def steps(lo, hi):
                for i in range(lo, hi):
                    run_step(PROG[c][i])

            def main():
                steps(1, SPLIT[c])
                assert not vals, vals

            def tail():
                steps(SPLIT[c], len(PROG[c]))
                for it in list(ldesc) + list(recv_of[c]):
                    wait_item(it)
                if c != 2:
                    need_peer(2)
                for i, k in enumerate(POOLS):
                    if nsent[c][k]:
                        r = pool[k].at[pl.ds(0, nsent[c][k])]
                        pltpu.make_async_copy(r, r, ssem.at[i]).wait()

            def replayable(fn):
                state = (waited, known, staged, consumed, ldesc, vals, lazy, pstate)
                snap = []

                def run():
                    if not snap:
                        snap.append(([type(a)(a) for a in state], nl[0]))
                    for a, old in zip(state, snap[0][0]):
                        a.clear()
                        a.update(old)
                    nl[0] = snap[0][1]
                    fn()
                return run

            return [replayable(fn) for fn in (prologue, main, tail)]

        progs = [program(c) for c in range(4)]
        for phase in range(3):
            mark[0] = phase
            lax.cond(me == 1, progs[1][phase],
                     lambda: lax.cond(me == 3, progs[3][phase],
                                      lambda: lax.cond(me == 2, progs[2][phase], progs[0][phase])))

    def kernel(x, Wq, K_ext, V_ext, Wo):
        kt = K_ext.transpose(0, 2, 3, 1).reshape(2, 1024, 256)
        vt = V_ext.transpose(0, 2, 3, 1).reshape(2, 1024, 256)
        V = pltpu.VMEM
        scratch = [
            V((2, 256, 512), F32), V((512, 256), F32), V((2, 1024, 256), F32), V((2, 1024, 256), F32),
            V((256, 512), F32), V((256, 512), BF16), V((4, 128, 512), F32),
            V((nsl["t"], 128, 128), BF16), V((nsl["h"], 64, 128), BF16),
            V((nsl["l2"], 2, 128), F32), V((nsl["l1"], 1, 128), F32), V((nsl["ar"], 16, CW), BF16),
            pltpu.SemaphoreType.DMA((len(POOLS),)), pltpu.SemaphoreType.DMA((max(nrecv),)),
            pltpu.SemaphoreType.DMA((nload,)), pltpu.SemaphoreType.REGULAR, pltpu.SMEM((1,), jnp.int32),
        ]
        base = dict(collective_id=0, vmem_limit_bytes=64 * 1024 * 1024)
        try:
            params = pltpu.CompilerParams(**base, disable_semaphore_checks=True,
                                          fuse_transposed_lhs_in_matmul=True)
        except TypeError:
            params = pltpu.CompilerParams(**base)
        return pl.pallas_call(
            body,
            out_shape=jax.ShapeDtypeStruct((2, 256, 512), F32),
            in_specs=[pl.BlockSpec(memory_space=pl.ANY)] * 5,
            out_specs=pl.BlockSpec(memory_space=pltpu.VMEM),
            scratch_shapes=scratch,
            compiler_params=params,
        )(x, Wq, kt, vt, Wo)

    return kernel


_NCH = 16
_SPLIT = [30, 38, 38, 46]
_PROG_TEXT = """
# chip 0
l raw_wo_b1 ; l raw_k_0b0 ; l raw_wo_b0 ; l raw_k_2b0
c cvt wob1 < raw_wo_b1 > wob1
l raw_v_0b0 ; l raw_wo_a1 ; l raw_v_2a0 ; l raw_wo_a0 ; l raw_v_2b0 ; l raw_x_L1 ; l raw_wq_a ; l raw_k_2a0 ; l raw_wq_b ; c cvt wob0 < raw_wo_b0 > wob0
c cvt woa1 < raw_wo_a1 > woa1
l raw_x_L0 ; c vprep 2a0 < raw_v_2a0 > v0_2a0_0 v0_2a0_1 ; c kprep 2b0 < raw_k_2b0 > k0_2b0_0 k0_2b0_1
c cvt woa0 < raw_wo_a0 > woa0
s v0_2a0_1 1 v0_2a0_1
l raw_k_3b0 ; l raw_x_H0 ; l raw_k_0a0 ; l raw_v_0a0 ; s k0_2b0_1 3 k0_2b0_1 ; s v0_2a0_0 1 v0_2a0_0 ; s k0_2b0_0 3 k0_2b0_0
l raw_k_1b0 ; l raw_k_1a0 ; l raw_k_2b1 ; l raw_v_1a0 ; c vprep 2b0 < raw_v_2b0 > v0_2b0_0 v0_2b0_1 ; c kprep 0b0 < raw_k_0b0 > k0_0b0_0 k0_0b0_1 ; c kprep 2a0 < raw_k_2a0 > k0_2a0_0 k0_2a0_1 ; s k0_2a0_0 1 k0_2a0_0 ; s v0_2b0_1 3 v0_2b0_1 ; s k0_2a0_1 1 k0_2a0_1 ; s v0_2b0_0 3 v0_2b0_0
l raw_k_1b1 ; l raw_k_3a1 ; l raw_v_0b1 ; l raw_v_1b0 ; c qproj 0aL0 < raw_x_L0 raw_wq_a > q0aL0 ; c qproj 0aL1 < raw_x_L1 raw_wq_a > q0aL1 ; c qproj 0bL0 < raw_x_L0 raw_wq_b > q0bL0 ; c qproj 0bL1 < raw_x_L1 raw_wq_b > q0bL1
l raw_v_3b0 ; l raw_v_1b1 ; c qproj 0bH0 < raw_x_H0 raw_wq_b > q0bH0 ; c att0 0bL0 < q0bL0 k0_0b0_0 k0_0b0_1 raw_v_0b0 > c0_0bL0 ; c cq 00 < q0aL0 q0bL0 > cq00 ; c kprep 0a0 < raw_k_0a0 > k0_0a0_0 k0_0a0_1 ; c kprep 3b0 < raw_k_3b0 > k0_3b0_0 k0_3b0_1 ; c cq 01 < q0aL1 q0bL1 > cq01 ; s q0bH0 1 q0bH0 ; s cq01 3 cq01
l raw_v_1a1 ; l raw_k_3a0 ; c att0 0aL0 < q0aL0 k0_0a0_0 k0_0a0_1 raw_v_0a0 > c0_0aL0 ; s cq00 3 cq00
l raw_k_1a1 ; l raw_k_0b1 ; l raw_v_3a0 ; c proj 0aL0 < c0_0aL0 woa0 woa1 > ppL0_a ; c proj 0bL0 < c0_0bL0 wob0 wob1 > ppL0_b ; c kprep 1a0 < raw_k_1a0 > k0_1a0_0 k0_1a0_1 ; c kprep 1b0 < raw_k_1b0 > k0_1b0_0 k0_1b0_1 ; c kprep 2b1 < raw_k_2b1 > k0_2b1_0 k0_2b1_1 ; c pfin L0 < ppL0_a ppL0_b > PL0_4_0 PL0_5_0 PL0_6_0 PL0_7_0 PL0_8_0 PL0_9_0 PL0_10_0 PL0_11_0 PL0_12_0 PL0_13_0 PL0_14_0 PL0_15_0 ; s PL0_13_0 1 SL0_13_0@1r ; s PL0_5_0 3 SL0_5_0@3r ; s PL0_6_0 1 SL0_6_0@1r ; s PL0_12_0 3 SL0_12_0@3r
l raw_k_3b1 ; l raw_x_H1 ; c att0 1aL0 < q1aL0 k0_1a0_0 k0_1a0_1 raw_v_1a0 > c0_1aL0 ; c kprep 1b1 < raw_k_1b1 > k0_1b1_0 k0_1b1_1 ; s c0_1aL0 1 c0_1aL0 ; s PL0_9_0 3 SL0_9_0@3r ; s PL0_11_0 3 SL0_11_0@3r ; s PL0_4_0 3 SL0_4_0@3r ; s PL0_8_0 3 SL0_8_0@3r
l raw_v_3a1 ; l raw_k_0a1 ; l raw_v_2b1 ; c att0 1bL0 < q1bL0 k0_1b0_0 k0_1b0_1 raw_v_1b0 > c0_1bL0 ; c att0 3bL0 < q3bL0 k0_3b0_0 k0_3b0_1 raw_v_3b0 > c0_3bL0 ; s c0_1bL0 1 c0_1bL0 ; s c0_3bL0 3 c0_3bL0
l raw_v_2a1 ; l raw_v_3b1 ; l raw_k_2a1 ; c att0 0bH0 < q0bH0 k0_0b0_0 k0_0b0_1 raw_v_0b0 > c0_0bH0 ; c att0 1bL1 < q1bL1 k0_1b1_0 k0_1b1_1 raw_v_1b1 > c0_1bL1 ; c qproj 3aL0 < raw_x_L0 w3_a0 w3_a1 w3_a2 w3_a3 > q3aL0 ; c kprep 3a0 < raw_k_3a0 > k0_3a0_0 k0_3a0_1 ; s c0_1bL1 1 c0_1bL1 ; s PL0_14_0 3 SL0_14_0@3r
l raw_v_0a1 ; c qproj 0aH0 < raw_x_H0 raw_wq_a > q0aH0 ; c att0 3aL0 < q3aL0 k0_3a0_0 k0_3a0_1 raw_v_3a0 > c0_3aL0 ; c kprep 1a1 < raw_k_1a1 > k0_1a1_0 k0_1a1_1 ; s c0_3aL0 3 c0_3aL0
c att0 1aL1 < q1aL1 k0_1a1_0 k0_1a1_1 raw_v_1a1 > c0_1aL1 ; c qproj 3aH0 < raw_x_H0 w3_a0 w3_a1 w3_a2 w3_a3 > q3aH0 ; c kprep 0b1 < raw_k_0b1 > k0_0b1_0 k0_0b1_1 ; s c0_1aL1 1 c0_1aL1
c qproj 3aL1 < raw_x_L1 w3_a0 w3_a1 w3_a2 w3_a3 > q3aL1 ; c att0 3bH0 < q3bH0 k0_3b0_0 k0_3b0_1 raw_v_3b0 > c0_3bH0 ; s c0_3bH0 3 c0_3bH0
c att0 0bL1 < q0bL1 k0_0b1_0 k0_0b1_1 raw_v_0b1 > c0_0bL1 ; c att0 1aH0 < q1aH0 k0_1a0_0 k0_1a0_1 raw_v_1a0 > c0_1aH0 ; c att0 3aH0 < q3aH0 k0_3a0_0 k0_3a0_1 raw_v_3a0 > c0_3aH0 ; c kprep 0a1 < raw_k_0a1 > k0_0a1_0 k0_0a1_1 ; c kprep 3a1 < raw_k_3a1 > k0_3a1_0 k0_3a1_1 ; s c0_1aH0 1 c0_1aH0 ; s c0_3aH0 3 c0_3aH0
c qproj 0bH1 < raw_x_H1 raw_wq_b > q0bH1 ; c att0 1bH0 < q1bH0 k0_1b0_0 k0_1b0_1 raw_v_1b0 > c0_1bH0 ; c att0 2bL1 < q2bL1 k0_2b1_0 k0_2b1_1 raw_v_2b1 > c0_2bL1 ; c att0 3aL1 < q3aL1 k0_3a1_0 k0_3a1_1 raw_v_3a1 > c0_3aL1 ; c kprep 2a1 < raw_k_2a1 > k0_2a1_0 k0_2a1_1 ; s c0_1bH0 1 c0_1bH0 ; s c0_2bL1 2 c0_2bL1 ; s q0bH1 1 q0bH1 ; s c0_3aL1 3 c0_3aL1
c att0 0aL1 < q0aL1 k0_0a1_0 k0_0a1_1 raw_v_0a1 > c0_0aL1 ; c att0 1bH1 < q1bH1 k0_1b1_0 k0_1b1_1 raw_v_1b1 > c0_1bH1 ; c att0 2aH1 < q2aH1 k0_2a1_0 k0_2a1_1 raw_v_2a1 > c0_2aH1 ; c att0 2aL1 < q2aL1 k0_2a1_0 k0_2a1_1 raw_v_2a1 > c0_2aL1 ; c kprep 3b1 < raw_k_3b1 > k0_3b1_0 k0_3b1_1 ; s c0_2aH1 1 c0_2aH1 ; s c0_2aL1 2 c0_2aL1
c qproj 0aH1 < raw_x_H1 raw_wq_a > q0aH1 ; c proj 0aL1 < c0_0aL1 woa0 woa1 > ppL1_a ; c att0 0bH1 < q0bH1 k0_0b1_0 k0_0b1_1 raw_v_0b1 > c0_0bH1 ; c att0 2bH1 < q2bH1 k0_2b1_0 k0_2b1_1 raw_v_2b1 > c0_2bH1 ; c att0 3bL1 < q3bL1 k0_3b1_0 k0_3b1_1 raw_v_3b1 > c0_3bL1 ; s c0_2bH1 1 c0_2bH1 ; s c0_3bL1 3 c0_3bL1
c proj 0bL1 < c0_0bL1 wob0 wob1 > ppL1_b ; c qproj 3aH1 < raw_x_H1 w3_a0 w3_a1 w3_a2 w3_a3 > q3aH1 ; c att0 3bH1 < q3bH1 k0_3b1_0 k0_3b1_1 raw_v_3b1 > c0_3bH1
c merge 3bH1 < c0_3bH1 c1_3bH1 > m_3bH1 ; c add L0.7 03@0 < PL0_7_0 SL0_7_3@0r > SL0_7_03@0 ; c pfin L1 < ppL1_a ppL1_b > PL1_4_0 PL1_5_0 PL1_6_0 PL1_7_0 PL1_8_0 PL1_9_0 PL1_10_0 PL1_11_0 PL1_12_0 PL1_13_0 PL1_14_0 PL1_15_0 ; s PL1_8_0 1 SL1_8_0@1r
c att0 3aH1 < q3aH1 k0_3a1_0 k0_3a1_1 raw_v_3a1 > c0_3aH1
c out L0.4 < SL0_4_0123@0r > outL04 ; s c0_1bH1 1 c0_1bH1 ; s PL1_14_0 3 SL1_14_0@3r ; s m_3bH1 3 m_3bH1
c att01 0aH0 < q0aH0 k0_0a0_0 k0_0a0_1 raw_v_0a0 k1_0a0_0 v1_0a0_0 > c0_0aH0 ; c att0 1aH1 < q1aH1 k0_1a1_0 k0_1a1_1 raw_v_1a1 > c0_1aH1 ; s PL1_5_0 1 SL1_5_0@1r
c proj 0aH0 < c0_0aH0 woa0 woa1 > ppH0_a ; c att01 0aH1 < q0aH1 k0_0a1_0 k0_0a1_1 raw_v_0a1 k1_0a1_0 v1_0a1_0 > c0_0aH1
c merge 3aH1 < c0_3aH1 c1_3aH1 > m_3aH1 ; s c0_1aH1 1 c0_1aH1 ; s m_3aH1 3 m_3aH1
c add L0.11 0123@0 < SL0_11_123@0r PL0_11_0 > SL0_11_0123@0 ; c out L0.11 < SL0_11_0123@0 > outL011 ; s PL1_6_0 1 SL1_6_0@1r ; s PL1_10_0 3 SL1_10_0@3r ; s PL1_13_0 1 SL1_13_0@1r
c zmerge 0bH0 < c0_0bH0 c1_0bH0 > m_0bH0 ; c proj 0bH0 < m_0bH0 wob0 wob1 > ppH0_b
c out L0.5 < SL0_5_0123@0r > outL05 ; c pfin H0 < ppH0_a ppH0_b > PH0_0_0 PH0_1_0 PH0_2_0 PH0_3_0 PH0_4_0 PH0_5_0 PH0_6_0 PH0_7_0 PH0_8_0 PH0_9_0 PH0_10_0 PH0_11_0 PH0_12_0 PH0_13_0 PH0_14_0 PH0_15_0 ; c add H0.4 03@0 < PH0_4_0 SH0_4_3@0r > SH0_4_03@0 ; c add H0.9 03@0 < PH0_9_0 SH0_9_3@0r > SH0_9_03@0 ; s PH0_6_0 3 SH0_6_0@3r ; s SH0_4_03@0 1 SH0_4_03@1r
c out L0.9 < SL0_9_0123@0r > outL09 ; s PL1_7_0 3 SL1_7_0@3r ; s SH0_9_03@0 1 SH0_9_03@1r ; s PH0_15_0 3 SH0_15_0@3r
c out L0.12 < SL0_12_0123@0r > outL012 ; s PH0_13_0 1 SH0_13_0@1r ; s PH0_5_0 3 SH0_5_0@3r
c add L0.8 0123@0 < SL0_8_123@0r PL0_8_0 > SL0_8_0123@0 ; c out L0.8 < SL0_8_0123@0 > outL08 ; s PH0_11_0 1 SH0_11_0@1r ; s PL1_9_0 3 SL1_9_0@3r
c proj 0aH1 < c0_0aH1 woa0 woa1 > ppH1_a ; c zmerge 0bH1 < c0_0bH1 c1_0bH1 > m_0bH1 ; c proj 0bH1 < m_0bH1 wob0 wob1 > ppH1_b
c out L0.6 < SL0_6_0123@0r > outL06 ; c pfin H1 < ppH1_a ppH1_b > PH1_0_0 PH1_1_0 PH1_2_0 PH1_3_0 PH1_4_0 PH1_5_0 PH1_6_0 PH1_7_0 PH1_8_0 PH1_9_0 PH1_10_0 PH1_11_0 PH1_12_0 PH1_13_0 PH1_14_0 PH1_15_0 ; s PH1_10_0 1 SH1_10_0@1r ; s PH1_13_0 3 SH1_13_0@3r ; s PH1_3_0 1 SH1_3_0@1r ; s PH1_1_0 3 SH1_1_0@3r
c gfinal 00 < gacc00_3r gp00_1r > gm00 ; c pfing L0 < c0_0aL0 c0_0bL0 gm00 woa0 woa1 wob0 wob1 > PL0_0_0 PL0_1_0 PL0_2_0 PL0_3_0
c add L0.15 0123@0 < SL0_15_12@0r PL0_15_0 SL0_15_3@0r > SL0_15_0123@0 ; c add L0.10 01@0 < PL0_10_0 SL0_10_1@0r > SL0_10_01@0 ; c add L0.10 0123@0 < SL0_10_01@0 SL0_10_23@0r > SL0_10_0123@0 ; c out L0.15 < SL0_15_0123@0 > outL015 ; s PH1_12_0 1 SH1_12_0@1r
c out L0.10 < SL0_10_0123@0 > outL010 ; s PL0_3_0 3 SL0_3_0@3r
c out L0.14 < SL0_14_0123@0r > outL014 ; s PH1_14_0 1 SH1_14_0@1r ; s PH1_7_0 3 SH1_7_0@3r ; s PH1_4_0 1 SH1_4_0@1r ; s PL0_1_0 3 SL0_1_0@3r ; c out L0.13 < SL0_13_0123@0r > outL013
c add L1.4 03@0 < PL1_4_0 SL1_4_3@0r > SL1_4_03@0 ; s SL1_4_03@0 1 SL1_4_03@1r ; s PH1_8_0 3 SH1_8_0@3r
c gfinal 01 < gacc01_1r > gm01 ; c pfing L1 < c0_0aL1 c0_0bL1 gm01 woa0 woa1 wob0 wob1 > PL1_0_0 PL1_1_0 PL1_2_0 PL1_3_0
c add H0.10 0123@0 < SH0_10_23@0r PH0_10_0 SH0_10_1@0r > SH0_10_0123@0 ; c out H0.10 < SH0_10_0123@0 > outH010 ; s PL1_0_0 1 SL1_0_0@1r ; s PL1_2_0 3 SL1_2_0@3r ; s PH1_2_0 1 SH1_2_0@1r ; s PL1_1_0 3 SL1_1_0@3r
c add L1.12 03@0 < PL1_12_0 SL1_12_3@0r > SL1_12_03@0 ; s PL1_15_0 1 SL1_15_0@1r ; s PH1_0_0 3 SH1_0_0@3r
c add L0.2 0123@0 < SL0_2_23@0r PL0_2_0 SL0_2_1@0r > SL0_2_0123@0 ; c out L0.2 < SL0_2_0123@0 > outL02 ; c add H0.12 01@0 < PH0_12_0 SH0_12_1@0r > SH0_12_01@0 ; c add H0.12 0123@0 < SH0_12_01@0 SH0_12_23@0r > SH0_12_0123@0 ; c out H0.12 < SH0_12_0123@0 > outH012 ; s PH0_3_0 1 SH0_3_0@1r ; s PH1_11_0 3 SH1_11_0@3r
c add H0.5 0123@0 < SH0_5_123@0r PH0_5_0 > SH0_5_0123@0 ; c out H0.5 < SH0_5_0123@0 > outH05 ; c add H0.7 01@0 < PH0_7_0 SH0_7_1@0r > SH0_7_01@0 ; c add H0.7 0123@0 < SH0_7_01@0 SH0_7_23@0r > SH0_7_0123@0 ; c out H0.7 < SH0_7_0123@0 > outH07 ; s SL0_7_03@0 1 SL0_7_03@1r ; s PH0_1_0 3 SH0_1_0@3r
c add H0.0 0123@0 < SH0_0_123@0r PH0_0_0 > SH0_0_0123@0 ; c out H0.0 < SH0_0_0123@0 > outH00 ; c add H0.2 0123@0 < SH0_2_23@0r PH0_2_0 SH0_2_1@0r > SH0_2_0123@0 ; c out H0.2 < SH0_2_0123@0 > outH02 ; s PL1_3_0 1 SL1_3_0@1r ; s SL0_15_0123@0 3 SL0_15_0123@3r
c add H1.15 03@0 < PH1_15_0 SH1_15_3@0r > SH1_15_03@0 ; c add H0.8 0123@0 < SH0_8_23@0r PH0_8_0 SH0_8_1@0r > SH0_8_0123@0 ; c out H0.8 < SH0_8_0123@0 > outH08 ; s SH0_2_0123@0 1 SH0_2_0123@1r ; s PH1_6_0 3 SH1_6_0@3r
c add H0.1 0123@0 < SH0_1_123@0r PH0_1_0 > SH0_1_0123@0 ; c add L0.0 0123@0 < SL0_0_12@0r PL0_0_0 SL0_0_3@0r > SL0_0_0123@0 ; c out H0.1 < SH0_1_0123@0 > outH01 ; c out L0.0 < SL0_0_0123@0 > outL00 ; s SH1_15_03@0 1 SH1_15_03@1r ; s PH0_0_0 3 SH0_0_0@3r
c out H0.6 < SH0_6_0123@0r > outH06 ; s SH0_12_0123@0 1 SH0_12_0123@1r ; s PH1_9_0 3 SH1_9_0@3r
c add L1.9 0123@0 < SL1_9_123@0r PL1_9_0 > SL1_9_0123@0 ; c add H0.14 01@0 < PH0_14_0 SH0_14_1@0r > SH0_14_01@0 ; c out L1.9 < SL1_9_0123@0 > outL19 ; c add H0.14 0123@0 < SH0_14_01@0 SH0_14_23@0r > SH0_14_0123@0 ; c out H0.14 < SH0_14_0123@0 > outH014 ; s SH0_10_0123@0 1 SH0_10_0123@1r ; s SH0_12_01@0 3 SH0_12_01@3r
c out H0.15 < SH0_15_0123@0r > outH015 ; c out H0.4 < SH0_4_0123@0r > outH04 ; s SL0_15_0123@0 1 SL0_15_0123@1r ; s SH0_14_01@0 3 SH0_14_01@3r
c out L1.7 < SL1_7_0123@0r > outL17 ; c add L1.12 0123@0 < SL1_12_03@0 SL1_12_12@0r > SL1_12_0123@0 ; c out L1.12 < SL1_12_0123@0 > outL112 ; s SL0_2_0123@0 1 SL0_2_0123@1r ; s SL0_10_01@0 3 SL0_10_01@3r
c add L1.14 0123@0 < SL1_14_123@0r PL1_14_0 > SL1_14_0123@0 ; c out H0.9 < SH0_9_0123@0r > outH09 ; c out L1.14 < SL1_14_0123@0 > outL114 ; s SH0_7_0123@0 1 SH0_7_0123@1r ; s SH0_2_0123@0 3 SH0_2_0123@3r
c out L1.10 < SL1_10_0123@0r > outL110 ; c add L1.11 0123@0 < SL1_11_12@0r PL1_11_0 SL1_11_3@0r > SL1_11_0123@0 ; c out L1.11 < SL1_11_0123@0 > outL111 ; s SL0_0_0123@0 1 SL0_0_0123@1r ; s SH0_10_0123@0 3 SH0_10_0123@3r
c out L0.3 < SL0_3_0123@0r > outL03 ; c out H0.13 < SH0_13_0123@0r > outH013 ; s SL0_10_0123@0 1 SL0_10_0123@1r ; s SL0_0_0123@0 3 SL0_0_0123@3r
c out L1.8 < SL1_8_0123@0r > outL18 ; c add H0.3 0123@0 < SH0_3_123@0r PH0_3_0 > SH0_3_0123@0 ; c out H0.3 < SH0_3_0123@0 > outH03 ; s SL1_12_03@0 1 SL1_12_03@1r ; s SH0_7_01@0 3 SH0_7_01@3r
c out L0.1 < SL0_1_0123@0r > outL01 ; c add H0.11 0123@0 < SH0_11_123@0r PH0_11_0 > SH0_11_0123@0 ; c out H0.11 < SH0_11_0123@0 > outH011 ; s SL1_7_0123@0r 1 SL1_7_0123@1r ; s SL0_2_0123@0 3 SL0_2_0123@3r
c add H1.5 0123@0 < SH1_5_23@0r PH1_5_0 SH1_5_1@0r > SH1_5_0123@0 ; c out H1.5 < SH1_5_0123@0 > outH15 ; c out L1.4 < SL1_4_0123@0r > outL14 ; s SH1_5_0123@0 1 SH1_5_0123@1r ; s SH1_5_0123@0 3 SH1_5_0123@3r
c out L1.2 < SL1_2_0123@0r > outL12 ; c out L1.6 < SL1_6_0123@0r > outL16 ; s SH0_8_0123@0 1 SH0_8_0123@1r ; s SL1_11_0123@0 3 SL1_11_0123@3r
c out L1.5 < SL1_5_0123@0r > outL15 ; c add H1.15 0123@0 < SH1_15_03@0 SH1_15_12@0r > SH1_15_0123@0 ; c out H1.15 < SH1_15_0123@0 > outH115 ; s SH0_14_0123@0 1 SH0_14_0123@1r ; s SH1_15_0123@0 3 SH1_15_0123@3r
c out L1.1 < SL1_1_0123@0r > outL11 ; c out L1.13 < SL1_13_0123@0r > outL113 ; s SH0_15_0123@0r 1 SH0_15_0123@1r ; s SL1_6_0123@0r 3 SL1_6_0123@3r
c out H1.8 < SH1_8_0123@0r > outH18 ; c out L1.15 < SL1_15_0123@0r > outL115 ; s SH1_8_0123@0r 1 SH1_8_0123@1r ; s SH0_8_0123@0 3 SH0_8_0123@3r
c add H1.6 0123@0 < SH1_6_123@0r PH1_6_0 > SH1_6_0123@0 ; c add L1.0 0123@0 < SL1_0_123@0r PL1_0_0 > SL1_0_0123@0 ; c out H1.6 < SH1_6_0123@0 > outH16 ; c out L1.0 < SL1_0_0123@0 > outL10 ; s SL1_11_0123@0 1 SL1_11_0123@1r ; s SL1_12_0123@0 3 SL1_12_0123@3r
c out H1.0 < SH1_0_0123@0r > outH10 ; c out L0.7 < SL0_7_0123@0r > outL07
c out H1.7 < SH1_7_0123@0r > outH17 ; s SH1_7_0123@0r 1 SH1_7_0123@1r ; c out L1.3 < SL1_3_0123@0r > outL13 ; s SL1_3_0123@0r 3 SL1_3_0123@3r
c add H1.1 0123@0 < SH1_1_123@0r PH1_1_0 > SH1_1_0123@0 ; c out H1.14 < SH1_14_0123@0r > outH114 ; c out H1.1 < SH1_1_0123@0 > outH11
c out H1.9 < SH1_9_0123@0r > outH19 ; c add H1.4 0123@0 < SH1_4_123@0r PH1_4_0 > SH1_4_0123@0 ; c out H1.4 < SH1_4_0123@0 > outH14
c out H1.11 < SH1_11_0123@0r > outH111 ; c out H1.2 < SH1_2_0123@0r > outH12
c out H1.13 < SH1_13_0123@0r > outH113 ; c add H1.12 0123@0 < SH1_12_123@0r PH1_12_0 > SH1_12_0123@0 ; c out H1.12 < SH1_12_0123@0 > outH112
c out H1.10 < SH1_10_0123@0r > outH110 ; c out H1.3 < SH1_3_0123@0r > outH13
# chip 1
l raw_v_0a0 ; l raw_wq_a ; l raw_x_L0
c vprep 0a0 < raw_v_0a0 > v1_0a0_0 ; s v1_0a0_0 0 v1_0a0_0
l raw_wq_b ; l raw_v_3b0 ; l raw_v_0b0 ; l raw_k_3b0 ; l raw_x_L1 ; l raw_k_0b0 ; l raw_k_2b0 ; l raw_v_2b0 ; l raw_x_H0 ; c qproj 1aL0 < raw_x_L0 raw_wq_a > q1aL0 ; s q1aL0 0 q1aL0
c qproj 1bL0 < raw_x_L0 raw_wq_b > q1bL0 ; s q1bL0 0 q1bL0
l raw_k_0b1 ; l raw_k_2a0 ; l raw_v_3b1 ; l raw_k_3a0 ; c vprep 3b0 < raw_v_3b0 > v1_3b0_0 ; c cq 10 < q1aL0 q1bL0 > cq10 ; s cq10 2 cq10 ; s v1_3b0_0 2 v1_3b0_0
l raw_wo_a1 ; l raw_v_2a0 ; c qproj 1aL1 < raw_x_L1 raw_wq_a > q1aL1 ; c qproj 1bL1 < raw_x_L1 raw_wq_b > q1bL1 ; s q1bL1 0 q1bL1
l raw_v_0b1 ; c kprep 3b0 < raw_k_3b0 > k1_3b0_0 ; c cq 11 < q1aL1 q1bL1 > cq11 ; s cq11 2 cq11 ; s k1_3b0_0 2 k1_3b0_0
l raw_x_H1 ; c kprep 2b0 < raw_k_2b0 > k1_2b0_0 ; s q1aL1 0 q1aL1
l raw_wo_b0 ; l raw_wo_b1 ; c qproj 1bH0 < raw_x_H0 raw_wq_b > q1bH0
l raw_k_0a0 ; l raw_v_2a1 ; l raw_v_3a0 ; c qproj 1aH0 < raw_x_H0 raw_wq_a > q1aH0 ; c att1 2bH0 < q2bH0 k1_2b0_0 raw_v_2b0 > c1_2bH0 ; c kprep 2a0 < raw_k_2a0 > k1_2a0_0 ; s c1_2bH0 2 c1_2bH0 ; s q1aH0 0 q1aH0
l raw_v_0a1 ; l raw_v_1a1 ; c cvt woa1 < raw_wo_a1 > woa1
l raw_k_3a1 ; l raw_k_3b1 ; c att01 2aH0 < q2aH0 k0_2a0_0 k0_2a0_1 v0_2a0_0 v0_2a0_1 k1_2a0_0 raw_v_2a0 > c0_2aH0 ; s c0_2aH0 2 c0_2aH0 ; s q1bH0 0 q1bH0
l raw_k_1a0 ; c kprep 0b0 < raw_k_0b0 > k1_0b0_0
c cvt wob0 < raw_wo_b0 > wob0
l raw_wo_a0 ; l raw_k_2a1 ; c qproj 1bH1 < raw_x_H1 raw_wq_b > q1bH1 ; c att0 2aL0 < q2aL0 k0_2a0_0 k0_2a0_1 v0_2a0_0 v0_2a0_1 > c0_2aL0 ; c kprep 3a0 < raw_k_3a0 > k1_3a0_0 ; c kprep 0b1 < raw_k_0b1 > k1_0b1_0
l raw_k_0a1 ; l raw_v_1a0 ; l raw_k_1b0 ; c cvt wob1 < raw_wo_b1 > wob1 ; s q1bH1 0 q1bH1 ; s c0_2aL0 2 c0_2aL0
l raw_k_2b1 ; l raw_v_3a1 ; l raw_v_2b1 ; c vprep 0a1 < raw_v_0a1 > v1_0a1_0 ; c qproj 1aH1 < raw_x_H1 raw_wq_a > q1aH1 ; c att1 3aH0 < q3aH0 k1_3a0_0 raw_v_3a0 > c1_3aH0 ; s c1_3aH0 3 c1_3aH0 ; s v1_0a1_0 0 v1_0a1_0
l raw_v_1b1 ; l raw_k_1a1 ; l raw_k_1b1 ; c kprep 0a0 < raw_k_0a0 > k1_0a0_0 ; c gatt 20 < cq20 raw_k_2a0 raw_k_2b0 raw_v_2a0 raw_v_2b0 > gp20_1 ; c kprep 3b1 < raw_k_3b1 > k1_3b1_0
c cvt woa0 < raw_wo_a0 > woa0 ; s gp20_1 2 gp20_1r ; s q1aH1 0 q1aH1
l raw_v_1b0 ; c proj 1aL0 < c0_1aL0 woa0 woa1 > ppL0_a ; c proj 1bL0 < c0_1bL0 wob0 wob1 > ppL0_b ; c kprep 1a0 < raw_k_1a0 > k1_1a0_0 ; c pfin L0 < ppL0_a ppL0_b > PL0_4_1 PL0_5_1 PL0_6_1 PL0_7_1 PL0_8_1 PL0_9_1 PL0_10_1 PL0_11_1 PL0_12_1 PL0_13_1 PL0_14_1 PL0_15_1 ; c add L0.13 01@1 < PL0_13_1 SL0_13_0@1r > SL0_13_01@1 ; c add L0.6 01@1 < PL0_6_1 SL0_6_0@1r > SL0_6_01@1 ; s PL0_4_1 3 SL0_4_1@3r ; s PL0_11_1 2 SL0_11_1@2r ; s PL0_5_1 2 SL0_5_1@2r ; s k1_0a0_0 0 k1_0a0_0 ; s PL0_8_1 2 SL0_8_1@2r
c proj 1bL1 < c0_1bL1 wob0 wob1 > ppL1_b ; c att1 3bH1 < q3bH1 k1_3b1_0 raw_v_3b1 > c1_3bH1 ; c kprep 1b0 < raw_k_1b0 > k1_1b0_0 ; c kprep 3a1 < raw_k_3a1 > k1_3a1_0 ; s PL0_12_1 2 SL0_12_1@2r ; s PL0_9_1 2 SL0_9_1@2r ; s SL0_13_01@1 2 SL0_13_01@2r ; s c1_3bH1 0 c1_3bH1 ; s PL0_14_1 2 SL0_14_1@2r ; s SL0_6_01@1 2 SL0_6_01@2r
c att1 0bH0 < q0bH0 k1_0b0_0 raw_v_0b0 > c1_0bH0 ; c proj 1aL1 < c0_1aL1 woa0 woa1 > ppL1_a ; c att1 3aH1 < q3aH1 k1_3a1_0 raw_v_3a1 > c1_3aH1 ; c gatt 30 < cq30 raw_k_3a0 raw_k_3b0 raw_v_3a0 raw_v_3b0 > gp30_1 ; c kprep 0a1 < raw_k_0a1 > k1_0a1_0 ; s gp30_1 2 gp30_1r ; s k1_0a1_0 0 k1_0a1_0 ; c pfin L1 < ppL1_a ppL1_b > PL1_4_1 PL1_5_1 PL1_6_1 PL1_7_1 PL1_8_1 PL1_9_1 PL1_10_1 PL1_11_1 PL1_12_1 PL1_13_1 PL1_14_1 PL1_15_1 ; s PL1_10_1 2 SL1_10_1@2r ; s PL1_14_1 2 SL1_14_1@2r
c att1 1aH0 < q1aH0 k1_1a0_0 raw_v_1a0 > c1_1aH0 ; c att1 1bH0 < q1bH0 k1_1b0_0 raw_v_1b0 > c1_1bH0 ; c gatt 10 < cq10 raw_k_1a0 raw_k_1b0 raw_v_1a0 raw_v_1b0 > gp10_1 ; c kprep 1a1 < raw_k_1a1 > k1_1a1_0 ; c kprep 2a1 < raw_k_2a1 > k1_2a1_0 ; c kprep 2b1 < raw_k_2b1 > k1_2b1_0 ; c gatt 31 < cq31 raw_k_3a1 raw_k_3b1 raw_v_3a1 raw_v_3b1 > gp31_1 ; s gp31_1 2 gp31_1r ; s c1_3aH1 0 c1_3aH1 ; s PL1_7_1 2 SL1_7_1@2r ; s PL1_9_1 2 SL1_9_1@2r
c zmerge 1aH0 < c0_1aH0 c1_1aH0 > m_1aH0 ; c proj 1aH0 < m_1aH0 woa0 woa1 > ppH0_a ; c att1 1aH1 < q1aH1 k1_1a1_0 raw_v_1a1 > c1_1aH1 ; c zmerge 1bH0 < c0_1bH0 c1_1bH0 > m_1bH0 ; c proj 1bH0 < m_1bH0 wob0 wob1 > ppH0_b ; c pfin H0 < ppH0_a ppH0_b > PH0_0_1 PH0_1_1 PH0_2_1 PH0_3_1 PH0_4_1 PH0_5_1 PH0_6_1 PH0_7_1 PH0_8_1 PH0_9_1 PH0_10_1 PH0_11_1 PH0_12_1 PH0_13_1 PH0_14_1 PH0_15_1 ; s PH0_15_1 2 SH0_15_1@2r ; s PH0_5_1 2 SH0_5_1@2r ; s c1_0bH0 0 c1_0bH0 ; s PH0_0_1 2 SH0_0_1@2r ; s PH0_6_1 2 SH0_6_1@2r ; s PH0_1_1 2 SH0_1_1@2r
c att1 0bH1 < q0bH1 k1_0b1_0 raw_v_0b1 > c1_0bH1 ; c gatt 00 < cq00 raw_k_0a0 raw_k_0b0 raw_v_0a0 raw_v_0b0 > gp00_1 ; c kprep 1b1 < raw_k_1b1 > k1_1b1_0 ; c gatt 21 < cq21 raw_k_2a1 raw_k_2b1 raw_v_2a1 raw_v_2b1 > gp21_1
c out L0.5 < SL0_5_0123@1r > outL05 ; s gp21_1 2 gp21_1r ; s c1_0bH1 0 c1_0bH1
c att1 2aH1 < q2aH1 k1_2a1_0 raw_v_2a1 > c1_2aH1 ; c att1 2bH1 < q2bH1 k1_2b1_0 raw_v_2b1 > c1_2bH1
c merge 2aH1 < c0_2aH1 c1_2aH1 > m_2aH1 ; s m_2aH1 2 m_2aH1 ; s gp00_1 0 gp00_1r
c gatt 01 < cq01 raw_k_0a1 raw_k_0b1 raw_v_0a1 raw_v_0b1 > gp01_1 ; c gatt 11 < cq11 raw_k_1a1 raw_k_1b1 raw_v_1a1 raw_v_1b1 > gp11_1 ; c add L0.15 12@1 < PL0_15_1 SL0_15_2@1r > SL0_15_12@1 ; s SL0_15_12@1 0 SL0_15_12@0r
c gmerge 01 < gp01_1 gacc01_2r > gacc01_1 ; c merge 2bH1 < c0_2bH1 c1_2bH1 > m_2bH1
c add L1.8 01@1 < PL1_8_1 SL1_8_0@1r > SL1_8_01@1 ; s SL1_8_01@1 2 SL1_8_01@2r ; s m_2bH1 2 m_2bH1 ; s PL0_10_1 0 SL0_10_1@0r
c att1 1bH1 < q1bH1 k1_1b1_0 raw_v_1b1 > c1_1bH1
c out L0.13 < SL0_13_0123@1r > outL013 ; s gacc01_1 0 gacc01_1r
c gfinal 10 < gp10_1 gacc10_2r > gm10 ; c pfing L0 < c0_1aL0 c0_1bL0 gm10 woa0 woa1 wob0 wob1 > PL0_0_1 PL0_1_1 PL0_2_1 PL0_3_1 ; c gfinal 11 < gp11_1 gacc11_2r > gm11 ; c pfing L1 < c0_1aL1 c0_1bL1 gm11 woa0 woa1 wob0 wob1 > PL1_0_1 PL1_1_1 PL1_2_1 PL1_3_1
c out L0.9 < SL0_9_0123@1r > outL09 ; c out L0.6 < SL0_6_0123@1r > outL06 ; c out L0.12 < SL0_12_0123@1r > outL012 ; s PH0_10_1 0 SH0_10_1@0r ; s PL1_2_1 2 SL1_2_1@2r
c add L1.5 01@1 < PL1_5_1 SL1_5_0@1r > SL1_5_01@1 ; s PL0_2_1 0 SL0_2_1@0r ; s PL0_3_1 3 SL0_3_1@3r
c zmerge 1bH1 < c0_1bH1 c1_1bH1 > m_1bH1 ; c proj 1bH1 < m_1bH1 wob0 wob1 > ppH1_b
c add L0.8 0123@1 < SL0_8_023@1r PL0_8_1 > SL0_8_0123@1 ; c out L0.8 < SL0_8_0123@1 > outL08 ; s PH0_12_1 0 SH0_12_1@0r ; s SL1_5_01@1 2 SL1_5_01@2r ; s PH0_7_1 0 SH0_7_1@0r ; s PL0_1_1 3 SL0_1_1@3r ; s PH0_2_1 0 SH0_2_1@0r ; s PL1_1_1 2 SL1_1_1@2r
c add L0.0 12@1 < PL0_0_1 SL0_0_2@1r > SL0_0_12@1 ; s PH0_8_1 0 SH0_8_1@0r
c out L0.4 < SL0_4_0123@1r > outL04
c zmerge 1aH1 < c0_1aH1 c1_1aH1 > m_1aH1 ; c proj 1aH1 < m_1aH1 woa0 woa1 > ppH1_a ; c pfin H1 < ppH1_a ppH1_b > PH1_0_1 PH1_1_1 PH1_2_1 PH1_3_1 PH1_4_1 PH1_5_1 PH1_6_1 PH1_7_1 PH1_8_1 PH1_9_1 PH1_10_1 PH1_11_1 PH1_12_1 PH1_13_1 PH1_14_1 PH1_15_1 ; s PH1_8_1 2 SH1_8_1@2r ; s SL0_0_12@1 0 SL0_0_12@0r
c add L0.11 0123@1 < SL0_11_023@1r PL0_11_1 > SL0_11_0123@1 ; c out L0.11 < SL0_11_0123@1 > outL011 ; s PH1_5_1 0 SH1_5_1@0r ; s PH1_6_1 2 SH1_6_1@2r ; s PH1_0_1 2 SH1_0_1@2r
c add L1.13 01@1 < PL1_13_1 SL1_13_0@1r > SL1_13_01@1 ; s PH0_14_1 0 SH0_14_1@0r ; s PH1_7_1 2 SH1_7_1@2r
c out L0.14 < SL0_14_0123@1r > outL014
c add H0.4 0123@1 < SH0_4_03@1r PH0_4_1 SH0_4_2@1r > SH0_4_0123@1 ; c out H0.4 < SH0_4_0123@1 > outH04 ; s SH0_4_0123@1 0 SH0_4_0123@0r ; s PH1_1_1 2 SH1_1_1@2r
c add L1.12 12@1 < PL1_12_1 SL1_12_2@1r > SL1_12_12@1
c add H0.9 0123@1 < SH0_9_03@1r PH0_9_1 SH0_9_2@1r > SH0_9_0123@1 ; c out H0.9 < SH0_9_0123@1 > outH09 ; s SL1_12_12@1 0 SL1_12_12@0r ; s PH1_9_1 2 SH1_9_1@2r
c add L1.11 12@1 < PL1_11_1 SL1_11_2@1r > SL1_11_12@1
c add H0.13 01@1 < PH0_13_1 SH0_13_0@1r > SH0_13_01@1 ; s SH0_9_0123@1 0 SH0_9_0123@0r ; s PH1_11_1 2 SH1_11_1@2r
c add H0.11 01@1 < PH0_11_1 SH0_11_0@1r > SH0_11_01@1 ; s SL1_11_12@1 0 SL1_11_12@0r ; s PH1_13_1 2 SH1_13_1@2r
c add H0.13 0123@1 < SH0_13_01@1 SH0_13_23@1r > SH0_13_0123@1 ; c out H0.13 < SH0_13_0123@1 > outH013
c add H1.10 01@1 < PH1_10_1 SH1_10_0@1r > SH1_10_01@1 ; s SH0_13_0123@1 0 SH0_13_0123@0r ; s SH1_10_01@1 2 SH1_10_01@2r
c add H0.3 123@1 < SH0_3_23@1r PH0_3_1 > SH0_3_123@1
c add H1.3 01@1 < PH1_3_1 SH1_3_0@1r > SH1_3_01@1 ; s SH0_3_123@1 0 SH0_3_123@0r ; s SH0_11_01@1 2 SH0_11_01@2r
c add H1.12 01@1 < PH1_12_1 SH1_12_0@1r > SH1_12_01@1 ; s SH1_12_01@1 2 SH1_12_01@2r
c add H0.11 123@1 < SH0_11_23@1r PH0_11_1 > SH0_11_123@1 ; c add H0.11 0123@1 < SH0_11_123@1 SH0_11_0@1r > SH0_11_0123@1 ; c out H0.11 < SH0_11_0123@1 > outH011 ; s SH0_11_123@1 0 SH0_11_123@0r
c add H1.14 01@1 < PH1_14_1 SH1_14_0@1r > SH1_14_01@1 ; s SH1_3_01@1 2 SH1_3_01@2r
c out L1.8 < SL1_8_0123@1r > outL18
c add H1.4 01@1 < PH1_4_1 SH1_4_0@1r > SH1_4_01@1 ; s SH0_13_01@1 2 SH0_13_01@2r
c add L1.14 0123@1 < SL1_14_023@1r PL1_14_1 > SL1_14_0123@1 ; c out L1.14 < SL1_14_0123@1 > outL114
c add L1.4 0123@1 < SL1_4_03@1r PL1_4_1 SL1_4_2@1r > SL1_4_0123@1 ; c out L1.4 < SL1_4_0123@1 > outL14 ; s SL1_4_0123@1 0 SL1_4_0123@0r ; s SH1_14_01@1 2 SH1_14_01@2r
c add L1.6 0123@1 < SL1_6_23@1r PL1_6_1 SL1_6_0@1r > SL1_6_0123@1 ; c out L1.6 < SL1_6_0123@1 > outL16 ; s SL1_6_0123@1 0 SL1_6_0123@0r
c add L1.0 01@1 < PL1_0_1 SL1_0_0@1r > SL1_0_01@1 ; s SL1_0_01@1 2 SL1_0_01@2r
c add H1.15 12@1 < PH1_15_1 SH1_15_2@1r > SH1_15_12@1 ; s SH1_15_12@1 0 SH1_15_12@0r
c add H1.2 01@1 < PH1_2_1 SH1_2_0@1r > SH1_2_01@1 ; s SL1_13_01@1 2 SL1_13_01@2r
c add L1.13 0123@1 < SL1_13_01@1 SL1_13_23@1r > SL1_13_0123@1 ; c out L1.13 < SL1_13_0123@1 > outL113 ; s SL1_13_0123@1 0 SL1_13_0123@0r
c add L1.15 01@1 < PL1_15_1 SL1_15_0@1r > SL1_15_01@1 ; c add L1.15 0123@1 < SL1_15_01@1 SL1_15_23@1r > SL1_15_0123@1 ; c out L1.15 < SL1_15_0123@1 > outL115 ; s SL1_15_0123@1 0 SL1_15_0123@0r ; s SH0_9_0123@1 2 SH0_9_0123@2r
c add L1.0 123@1 < SL1_0_23@1r PL1_0_1 > SL1_0_123@1 ; c add L1.0 0123@1 < SL1_0_123@1 SL1_0_0@1r > SL1_0_0123@1 ; c out L1.0 < SL1_0_0123@1 > outL10 ; s SL1_0_123@1 0 SL1_0_123@0r
c add H0.3 01@1 < PH0_3_1 SH0_3_0@1r > SH0_3_01@1 ; c add H0.3 0123@1 < SH0_3_123@1 SH0_3_0@1r > SH0_3_0123@1 ; c out H0.3 < SH0_3_0123@1 > outH03 ; s SH0_3_01@1 2 SH0_3_01@2r
c out L1.5 < SL1_5_0123@1r > outL15
c add L0.7 0123@1 < SL0_7_03@1r PL0_7_1 SL0_7_2@1r > SL0_7_0123@1 ; s SL0_7_0123@1 0 SL0_7_0123@0r ; c out L0.7 < SL0_7_0123@1 > outL07 ; s SH1_2_01@1 2 SH1_2_01@2r
c add L1.3 0123@1 < SL1_3_23@1r PL1_3_1 SL1_3_0@1r > SL1_3_0123@1 ; c out L1.3 < SL1_3_0123@1 > outL13 ; s SL1_3_0123@1 0 SL1_3_0123@0r ; s SH1_4_01@1 2 SH1_4_01@2r
c add H1.14 0123@1 < SH1_14_01@1 SH1_14_23@1r > SH1_14_0123@1 ; c out H1.14 < SH1_14_0123@1 > outH114 ; s SH1_14_0123@1 0 SH1_14_0123@0r
c out H0.2 < SH0_2_0123@1r > outH02 ; s SH0_4_0123@1 2 SH0_4_0123@2r
c add H1.4 123@1 < SH1_4_23@1r PH1_4_1 > SH1_4_123@1 ; c add H1.4 0123@1 < SH1_4_123@1 SH1_4_0@1r > SH1_4_0123@1 ; c out H1.4 < SH1_4_0123@1 > outH14 ; s SH1_4_123@1 0 SH1_4_123@0r
c add H1.15 0123@1 < SH1_15_03@1r SH1_15_12@1 > SH1_15_0123@1 ; c out H1.15 < SH1_15_0123@1 > outH115 ; s SL0_7_0123@1 2 SL0_7_0123@2r
c add H1.2 0123@1 < SH1_2_01@1 SH1_2_23@1r > SH1_2_0123@1 ; c out H1.2 < SH1_2_0123@1 > outH12 ; s SH1_2_0123@1 0 SH1_2_0123@0r
c out H0.12 < SH0_12_0123@1r > outH012 ; s SL1_4_0123@1 2 SL1_4_0123@2r
c out H0.6 < SH0_6_0123@1r > outH06
c out H0.10 < SH0_10_0123@1r > outH010 ; s SL1_15_01@1 2 SL1_15_01@2r
c add H1.12 123@1 < SH1_12_23@1r PH1_12_1 > SH1_12_123@1 ; c add H1.12 0123@1 < SH1_12_123@1 SH1_12_0@1r > SH1_12_0123@1 ; c out H1.12 < SH1_12_0123@1 > outH112 ; s SH1_12_123@1 0 SH1_12_123@0r
c out L0.15 < SL0_15_0123@1r > outL015 ; s SH0_10_0123@1r 2 SH0_10_0123@2r
c add H1.3 0123@1 < SH1_3_01@1 SH1_3_23@1r > SH1_3_0123@1 ; c out H1.3 < SH1_3_0123@1 > outH13 ; s SH1_3_0123@1 0 SH1_3_0123@0r
c out L0.2 < SL0_2_0123@1r > outL02 ; s SH0_2_0123@1r 2 SH0_2_0123@2r
c out L1.10 < SL1_10_0123@1r > outL110
c out H0.7 < SH0_7_0123@1r > outH07 ; s SL1_6_0123@1 2 SL1_6_0123@2r
c out H1.13 < SH1_13_0123@1r > outH113
c out L0.0 < SL0_0_0123@1r > outL00 ; s SH1_15_0123@1 2 SH1_15_0123@2r
c out H1.10 < SH1_10_0123@1r > outH110
c out L0.10 < SL0_10_0123@1r > outL010 ; s SL0_2_0123@1r 2 SL0_2_0123@2r
c add H1.1 0123@1 < SH1_1_023@1r PH1_1_1 > SH1_1_0123@1 ; c out H1.1 < SH1_1_0123@1 > outH11
c add L1.12 0123@1 < SL1_12_03@1r SL1_12_12@1 > SL1_12_0123@1 ; c out L1.12 < SL1_12_0123@1 > outL112 ; s SL1_3_0123@1 2 SL1_3_0123@2r
c add L1.9 0123@1 < SL1_9_023@1r PL1_9_1 > SL1_9_0123@1 ; c out L1.9 < SL1_9_0123@1 > outL19
c out L1.7 < SL1_7_0123@1r > outL17 ; s SL1_12_0123@1 2 SL1_12_0123@2r
c add H0.5 0123@1 < SH0_5_023@1r PH0_5_1 > SH0_5_0123@1 ; c out H0.5 < SH0_5_0123@1 > outH05
c out H1.5 < SH1_5_0123@1r > outH15 ; s SH1_5_0123@1r 2 SH1_5_0123@2r
c out L0.1 < SL0_1_0123@1r > outL01
c out H0.8 < SH0_8_0123@1r > outH08 ; s SH0_8_0123@1r 2 SH0_8_0123@2r
c out L0.3 < SL0_3_0123@1r > outL03
c out H0.14 < SH0_14_0123@1r > outH014
c out L1.2 < SL1_2_0123@1r > outL12
c out H0.15 < SH0_15_0123@1r > outH015
c out L1.1 < SL1_1_0123@1r > outL11
c out H1.8 < SH1_8_0123@1r > outH18
c out H1.0 < SH1_0_0123@1r > outH10
c out L1.11 < SL1_11_0123@1r > outL111
c out H1.11 < SH1_11_0123@1r > outH111
c out H1.7 < SH1_7_0123@1r > outH17
c add H0.1 0123@1 < SH0_1_023@1r PH0_1_1 > SH0_1_0123@1 ; c out H0.1 < SH0_1_0123@1 > outH01
c add H1.6 0123@1 < SH1_6_023@1r PH1_6_1 > SH1_6_0123@1 ; c out H1.6 < SH1_6_0123@1 > outH16
c add H0.0 0123@1 < SH0_0_023@1r PH0_0_1 > SH0_0_0123@1 ; c out H0.0 < SH0_0_0123@1 > outH00
c out H1.9 < SH1_9_0123@1r > outH19
# chip 2
l raw_wq_b2 ; l raw_wq_b1 ; l raw_wq_b3 ; l raw_wq_b0 ; l raw_x_H0
c cvtq 2b2 < raw_wq_b2 > w2_b2 ; s w2_b2 3 w2_b2
l raw_wo_b1 ; l raw_wo_b0 ; l raw_wq_a ; l raw_x_L1 ; l raw_x_L0 ; c cvtq 2b1 < raw_wq_b1 > w2_b1
c cvtq 2b3 < raw_wq_b3 > w2_b3
l raw_k_3b0 ; c cvtq 2b0 < raw_wq_b0 > w2_b0 ; s w2_b3 3 w2_b3
l raw_k_0b1 ; c qproj 2bH0 < raw_x_H0 w2_b0 w2_b1 w2_b2 w2_b3 > q2bH0 ; s q2bH0 1 q2bH0
l raw_x_H1 ; c cvt wob1 < raw_wo_b1 > wob1
l raw_k_0a0 ; c cvt wob0 < raw_wo_b0 > wob0 ; s w2_b1 3 w2_b1
l raw_wo_a1 ; l raw_v_0a0 ; l raw_k_2a0 ; l raw_v_0b0 ; c qproj 2aH0 < raw_x_H0 raw_wq_a > q2aH0 ; s q2aH0 1 q2aH0 ; s w2_b0 3 w2_b0
l raw_v_1b0 ; c qproj 2aL0 < raw_x_L0 raw_wq_a > q2aL0 ; s q2aL0 1 q2aL0
l raw_v_0a1 ; l raw_k_1a0 ; l raw_k_0a1 ; c qproj 2aL1 < raw_x_L1 raw_wq_a > q2aL1 ; c qproj 2bL0 < raw_x_L0 w2_b0 w2_b1 w2_b2 w2_b3 > q2bL0 ; s q2aL1 3 q2aL1 ; s q3aH0 1 q3aH0
c cq 20 < q2aL0 q2bL0 > cq20
l raw_k_0b0 ; l raw_wo_a0 ; c qproj 2aH1 < raw_x_H1 raw_wq_a > q2aH1 ; c qproj 2bL1 < raw_x_L1 w2_b0 w2_b1 w2_b2 w2_b3 > q2bL1
l raw_v_2b1 ; l raw_k_2b0 ; l raw_k_1a1 ; c cvt woa1 < raw_wo_a1 > woa1 ; s q2aH1 3 q2aH1 ; s cq20 1 cq20
l raw_v_2a1 ; l raw_k_2b1 ; s cq30 1 cq30 ; s cq10 3 cq10
l raw_v_3b0 ; l raw_v_0b1 ; s q3bH1 1 q3bH1 ; s cq11 3 cq11
l raw_k_1b1 ; l raw_v_3a0 ; c att1 3bH0 < q3bH0 k1_3b0_0 v1_3b0_0 > c1_3bH0 ; s cq20 3 cq20
c cvt woa0 < raw_wo_a0 > woa0
l raw_v_2a0 ; l raw_k_1b0 ; l raw_k_3a1 ; l raw_k_2a1 ; s q3aH1 1 q3aH1 ; s c1_3bH0 3 c1_3bH0
l raw_k_3a0 ; l raw_v_3b1 ; s cq31 1 cq31
l raw_v_2b0 ; s cq01 1 cq01
l raw_v_1a1 ; l raw_k_3b1 ; l raw_v_1b1 ; l raw_v_1a0 ; c gatt 00 < cq00 raw_k_0a0 raw_k_0b0 raw_v_0a0 raw_v_0b0 > gp00_2 ; s q2aH1 1 q2aH1 ; s gp00_2 3 gp00_2r ; s cq00 1 cq00
l raw_v_3a1 ; c proj 2aH0 < c0_2aH0 woa0 woa1 > ppH0_a ; c proj 2aL0 < c0_2aL0 woa0 woa1 > ppL0_a ; c proj 2bL0 < c0_2bL0 wob0 wob1 > ppL0_b ; c cq 21 < q2aL1 q2bL1 > cq21 ; c gatt 01 < cq01 raw_k_0a1 raw_k_0b1 raw_v_0a1 raw_v_0b1 > gp01_2 ; c pfin L0 < ppL0_a ppL0_b > PL0_4_2 PL0_5_2 PL0_6_2 PL0_7_2 PL0_8_2 PL0_9_2 PL0_10_2 PL0_11_2 PL0_12_2 PL0_13_2 PL0_14_2 PL0_15_2 ; s PL0_4_2 3 SL0_4_2@3r ; s PL0_10_2 3 SL0_10_2@3r ; s cq21 1 cq21
c zmerge 2bH0 < c0_2bH0 c1_2bH0 > m_2bH0 ; c proj 2bH0 < m_2bH0 wob0 wob1 > ppH0_b ; c qproj 2bH1 < raw_x_H1 w2_b0 w2_b1 w2_b2 w2_b3 > q2bH1 ; c pfin H0 < ppH0_a ppH0_b > PH0_0_2 PH0_1_2 PH0_2_2 PH0_3_2 PH0_4_2 PH0_5_2 PH0_6_2 PH0_7_2 PH0_8_2 PH0_9_2 PH0_10_2 PH0_11_2 PH0_12_2 PH0_13_2 PH0_14_2 PH0_15_2 ; s PH0_10_2 3 SH0_10_2@3r ; s PH0_8_2 3 SH0_8_2@3r
c gmerge 01 < gp01_2 gp01_3r > gacc01_2 ; s q2bH1 1 q2bH1 ; s PH0_12_2 3 SH0_12_2@3r ; s PH0_7_2 3 SH0_7_2@3r
c add L0.11 12@2 < PL0_11_2 SL0_11_1@2r > SL0_11_12@2 ; s SL0_11_12@2 3 SL0_11_12@3r ; s PH0_2_2 3 SH0_2_2@3r ; s PL0_7_2 1 SL0_7_2@1r
c gatt 30 < cq30 raw_k_3a0 raw_k_3b0 raw_v_3a0 raw_v_3b0 > gp30_2 ; c gatt 11 < cq11 raw_k_1a1 raw_k_1b1 raw_v_1a1 raw_v_1b1 > gp11_2 ; c gatt 21 < cq21 raw_k_2a1 raw_k_2b1 raw_v_2a1 raw_v_2b1 > gp21_2
c add L0.5 12@2 < PL0_5_2 SL0_5_1@2r > SL0_5_12@2 ; c add L0.5 0123@2 < SL0_5_03@2r SL0_5_12@2 > SL0_5_0123@2 ; c add L0.8 12@2 < PL0_8_2 SL0_8_1@2r > SL0_8_12@2 ; c add L0.12 12@2 < PL0_12_2 SL0_12_1@2r > SL0_12_12@2 ; c add L0.9 12@2 < PL0_9_2 SL0_9_1@2r > SL0_9_12@2 ; s SL0_5_12@2 3 SL0_5_12@3r
c gmerge 11 < gp11_2 gp11_3r > gacc11_2 ; s SL0_5_0123@2 1 SL0_5_0123@1r ; s SL0_9_12@2 3 SL0_9_12@3r ; s gacc01_2 1 gacc01_2r ; s SL0_12_12@2 3 SL0_12_12@3r
c out L0.5 < SL0_5_0123@2 > outL05 ; s SL0_8_12@2 3 SL0_8_12@3r ; s PL0_15_2 1 SL0_15_2@1r ; s PH0_14_2 3 SH0_14_2@3r ; s gacc11_2 1 gacc11_2r
c gatt 10 < cq10 raw_k_1a0 raw_k_1b0 raw_v_1a0 raw_v_1b0 > gp10_2 ; c gatt 20 < cq20 raw_k_2a0 raw_k_2b0 raw_v_2a0 raw_v_2b0 > gp20_2 ; c gatt 31 < cq31 raw_k_3a1 raw_k_3b1 raw_v_3a1 raw_v_3b1 > gp31_2
c add L0.12 0123@2 < SL0_12_03@2r SL0_12_12@2 > SL0_12_0123@2 ; c gmerge 10 < gp10_2 gp10_3r > gacc10_2 ; c add L0.6 0123@2 < SL0_6_01@2r PL0_6_2 SL0_6_3@2r > SL0_6_0123@2 ; c out L0.12 < SL0_12_0123@2 > outL012 ; s SL0_6_0123@2 3 SL0_6_0123@3r
c add L0.13 0123@2 < SL0_13_01@2r PL0_13_2 SL0_13_3@2r > SL0_13_0123@2 ; c add L0.14 12@2 < PL0_14_2 SL0_14_1@2r > SL0_14_12@2 ; c out L0.13 < SL0_13_0123@2 > outL013 ; c out L0.6 < SL0_6_0123@2 > outL06 ; s gacc10_2 1 gacc10_2r ; s SL0_14_12@2 3 SL0_14_12@3r ; s SL0_13_0123@2 3 SL0_13_0123@3r ; c gmerge 30 < gp30_2 gp30_1r > gacc30_2 ; s gacc30_2 3 gacc30_2r ; s SL0_13_0123@2 1 SL0_13_0123@1r
c gfinal 20 < gp20_2 gp20_1r gp20_3r > gm20 ; c pfing L0 < c0_2aL0 c0_2bL0 gm20 woa0 woa1 wob0 wob1 > PL0_0_2 PL0_1_2 PL0_2_2 PL0_3_2
c add L0.9 0123@2 < SL0_9_03@2r SL0_9_12@2 > SL0_9_0123@2 ; c gmerge 31 < gp31_2 gp31_1r > gacc31_2 ; s SL0_9_0123@2 1 SL0_9_0123@1r ; c out L0.9 < SL0_9_0123@2 > outL09 ; s SL0_6_0123@2 1 SL0_6_0123@1r ; s gacc31_2 3 gacc31_2r ; s SL0_12_0123@2 1 SL0_12_0123@1r ; s PL0_2_2 3 SL0_2_2@3r
c proj 2bL1 < c0_2bL1 wob0 wob1 > ppL1_b
c add L0.8 023@2 < SL0_8_03@2r PL0_8_2 > SL0_8_023@2 ; c add L0.8 0123@2 < SL0_8_023@2 SL0_8_1@2r > SL0_8_0123@2 ; c out L0.8 < SL0_8_0123@2 > outL08 ; s SL0_8_023@2 1 SL0_8_023@1r
c add H0.15 12@2 < PH0_15_2 SH0_15_1@2r > SH0_15_12@2 ; s PL0_3_2 3 SL0_3_2@3r ; s PH0_9_2 1 SH0_9_2@1r ; s PL0_1_2 3 SL0_1_2@3r ; s PL0_0_2 1 SL0_0_2@1r
c out L0.4 < SL0_4_0123@2r > outL04
c add H0.5 12@2 < PH0_5_2 SH0_5_1@2r > SH0_5_12@2 ; s SH0_5_12@2 3 SH0_5_12@3r ; s SL0_4_0123@2r 1 SL0_4_0123@1r
c add H0.0 12@2 < PH0_0_2 SH0_0_1@2r > SH0_0_12@2 ; s SH0_0_12@2 3 SH0_0_12@3r ; s PH0_4_2 1 SH0_4_2@1r
c add L0.11 023@2 < SL0_11_03@2r PL0_11_2 > SL0_11_023@2 ; c add L0.11 0123@2 < SL0_11_023@2 SL0_11_1@2r > SL0_11_0123@2 ; c out L0.11 < SL0_11_0123@2 > outL011
c add H0.6 12@2 < PH0_6_2 SH0_6_1@2r > SH0_6_12@2 ; s SH0_6_12@2 3 SH0_6_12@3r ; s SL0_11_023@2 1 SL0_11_023@1r
c add H0.1 12@2 < PH0_1_2 SH0_1_1@2r > SH0_1_12@2 ; s SH0_1_12@2 3 SH0_1_12@3r
c add L0.14 0123@2 < SL0_14_03@2r SL0_14_12@2 > SL0_14_0123@2 ; c out L0.14 < SL0_14_0123@2 > outL014 ; s SL0_14_0123@2 1 SL0_14_0123@1r ; s SH0_15_12@2 3 SH0_15_12@3r
c proj 2aL1 < c0_2aL1 woa0 woa1 > ppL1_a ; c pfin L1 < ppL1_a ppL1_b > PL1_4_2 PL1_5_2 PL1_6_2 PL1_7_2 PL1_8_2 PL1_9_2 PL1_10_2 PL1_11_2 PL1_12_2 PL1_13_2 PL1_14_2 PL1_15_2 ; s PL1_12_2 1 SL1_12_2@1r
c add L1.9 12@2 < PL1_9_2 SL1_9_1@2r > SL1_9_12@2 ; s SL1_9_12@2 3 SL1_9_12@3r
c add L1.7 12@2 < PL1_7_2 SL1_7_1@2r > SL1_7_12@2 ; c add L1.14 12@2 < PL1_14_2 SL1_14_1@2r > SL1_14_12@2 ; c add L1.10 12@2 < PL1_10_2 SL1_10_1@2r > SL1_10_12@2 ; c add H0.13 23@2 < PH0_13_2 SH0_13_3@2r > SH0_13_23@2 ; c add H0.3 23@2 < PH0_3_2 SH0_3_3@2r > SH0_3_23@2 ; s PL1_11_2 1 SL1_11_2@1r ; s SL1_7_12@2 3 SL1_7_12@3r ; s PL1_4_2 1 SL1_4_2@1r ; s SL1_14_12@2 3 SL1_14_12@3r ; s SH0_13_23@2 1 SH0_13_23@1r ; s SL1_10_12@2 3 SL1_10_12@3r ; s SH0_3_23@2 1 SH0_3_23@1r
c gfinal 21 < gp21_2 gp21_1r gp21_3r > gm21 ; c pfing L1 < c0_2aL1 c0_2bL1 gm21 woa0 woa1 wob0 wob1 > PL1_0_2 PL1_1_2 PL1_2_2 PL1_3_2
c add H0.11 23@2 < PH0_11_2 SH0_11_3@2r > SH0_11_23@2 ; c add L1.15 23@2 < PL1_15_2 SL1_15_3@2r > SL1_15_23@2 ; s SL1_15_23@2 1 SL1_15_23@1r ; s SH0_11_23@2 1 SH0_11_23@1r
c proj 2aH1 < m_2aH1 woa0 woa1 > ppH1_a
c add L1.8 0123@2 < SL1_8_01@2r PL1_8_2 SL1_8_3@2r > SL1_8_0123@2 ; c out L1.8 < SL1_8_0123@2 > outL18 ; s SL1_8_0123@2 3 SL1_8_0123@3r ; s SL1_8_0123@2 1 SL1_8_0123@1r
c add L1.14 023@2 < SL1_14_03@2r PL1_14_2 > SL1_14_023@2 ; c add L1.14 0123@2 < SL1_14_023@2 SL1_14_1@2r > SL1_14_0123@2 ; c out L1.14 < SL1_14_0123@2 > outL114 ; s SL1_14_023@2 1 SL1_14_023@1r
c add L1.6 23@2 < PL1_6_2 SL1_6_3@2r > SL1_6_23@2 ; s SL1_6_23@2 1 SL1_6_23@1r
c proj 2bH1 < m_2bH1 wob0 wob1 > ppH1_b ; c pfin H1 < ppH1_a ppH1_b > PH1_0_2 PH1_1_2 PH1_2_2 PH1_3_2 PH1_4_2 PH1_5_2 PH1_6_2 PH1_7_2 PH1_8_2 PH1_9_2 PH1_10_2 PH1_11_2 PH1_12_2 PH1_13_2 PH1_14_2 PH1_15_2 ; s PH1_5_2 3 SH1_5_2@3r
c add L1.2 12@2 < PL1_2_2 SL1_2_1@2r > SL1_2_12@2 ; s SL1_2_12@2 3 SL1_2_12@3r ; s PH1_15_2 1 SH1_15_2@1r
c add L1.13 23@2 < PL1_13_2 SL1_13_3@2r > SL1_13_23@2 ; s SL1_13_23@2 1 SL1_13_23@1r
c add L1.0 23@2 < PL1_0_2 SL1_0_3@2r > SL1_0_23@2 ; c add L1.5 0123@2 < SL1_5_01@2r PL1_5_2 SL1_5_3@2r > SL1_5_0123@2 ; c out L1.5 < SL1_5_0123@2 > outL15 ; s SL1_5_0123@2 3 SL1_5_0123@3r ; s SL1_0_23@2 1 SL1_0_23@1r ; s SL1_5_0123@2 1 SL1_5_0123@1r
c add L1.3 23@2 < PL1_3_2 SL1_3_3@2r > SL1_3_23@2 ; s SL1_3_23@2 1 SL1_3_23@1r
c add L1.1 12@2 < PL1_1_2 SL1_1_1@2r > SL1_1_12@2 ; s SL1_1_12@2 3 SL1_1_12@3r
c add H1.8 12@2 < PH1_8_2 SH1_8_1@2r > SH1_8_12@2 ; s SH1_8_12@2 3 SH1_8_12@3r
c add H1.14 23@2 < PH1_14_2 SH1_14_3@2r > SH1_14_23@2 ; s SH1_14_23@2 1 SH1_14_23@1r
c add H1.6 12@2 < PH1_6_2 SH1_6_1@2r > SH1_6_12@2 ; s SH1_6_12@2 3 SH1_6_12@3r
c add H1.4 23@2 < PH1_4_2 SH1_4_3@2r > SH1_4_23@2 ; s SH1_4_23@2 1 SH1_4_23@1r
c add H1.0 12@2 < PH1_0_2 SH1_0_1@2r > SH1_0_12@2 ; s SH1_0_12@2 3 SH1_0_12@3r
c add H1.2 23@2 < PH1_2_2 SH1_2_3@2r > SH1_2_23@2 ; s SH1_2_23@2 1 SH1_2_23@1r
c add H1.7 12@2 < PH1_7_2 SH1_7_1@2r > SH1_7_12@2 ; s SH1_7_12@2 3 SH1_7_12@3r
c add H0.6 0123@2 < SH0_6_03@2r SH0_6_12@2 > SH0_6_0123@2 ; c out H0.6 < SH0_6_0123@2 > outH06 ; s SH0_6_0123@2 1 SH0_6_0123@1r
c add H1.1 12@2 < PH1_1_2 SH1_1_1@2r > SH1_1_12@2 ; s SH1_1_12@2 3 SH1_1_12@3r
c add H1.12 23@2 < PH1_12_2 SH1_12_3@2r > SH1_12_23@2 ; s SH1_12_23@2 1 SH1_12_23@1r
c add H1.9 12@2 < PH1_9_2 SH1_9_1@2r > SH1_9_12@2 ; s SH1_9_12@2 3 SH1_9_12@3r
c add H1.3 23@2 < PH1_3_2 SH1_3_3@2r > SH1_3_23@2 ; s SH1_3_23@2 1 SH1_3_23@1r
c add H1.11 12@2 < PH1_11_2 SH1_11_1@2r > SH1_11_12@2 ; s SH1_11_12@2 3 SH1_11_12@3r
c add L1.10 0123@2 < SL1_10_03@2r SL1_10_12@2 > SL1_10_0123@2 ; c out L1.10 < SL1_10_0123@2 > outL110 ; s SL1_10_0123@2 1 SL1_10_0123@1r
c add H1.13 12@2 < PH1_13_2 SH1_13_1@2r > SH1_13_12@2 ; s SH1_13_12@2 3 SH1_13_12@3r
c add H1.10 0123@2 < SH1_10_01@2r PH1_10_2 SH1_10_3@2r > SH1_10_0123@2 ; s SH1_10_0123@2 3 SH1_10_0123@3r
c add H1.13 0123@2 < SH1_13_03@2r SH1_13_12@2 > SH1_13_0123@2 ; c out H1.13 < SH1_13_0123@2 > outH113 ; s SH1_13_0123@2 1 SH1_13_0123@1r ; c out H1.10 < SH1_10_0123@2 > outH110 ; s SH1_10_0123@2 1 SH1_10_0123@1r
c add H0.11 012@2 < SH0_11_01@2r PH0_11_2 > SH0_11_012@2 ; s SH0_11_012@2 3 SH0_11_012@3r
c add H1.1 023@2 < SH1_1_03@2r PH1_1_2 > SH1_1_023@2 ; c add H1.1 0123@2 < SH1_1_023@2 SH1_1_1@2r > SH1_1_0123@2 ; c out H1.1 < SH1_1_0123@2 > outH11 ; c add H0.11 0123@2 < SH0_11_012@2 SH0_11_3@2r > SH0_11_0123@2 ; c out H0.11 < SH0_11_0123@2 > outH011 ; s SH1_1_023@2 1 SH1_1_023@1r
c add H1.12 012@2 < SH1_12_01@2r PH1_12_2 > SH1_12_012@2 ; s SH1_12_012@2 3 SH1_12_012@3r
c add L1.9 023@2 < SL1_9_03@2r PL1_9_2 > SL1_9_023@2 ; c add L1.9 0123@2 < SL1_9_023@2 SL1_9_1@2r > SL1_9_0123@2 ; c add H1.12 0123@2 < SH1_12_012@2 SH1_12_3@2r > SH1_12_0123@2 ; c out L1.9 < SL1_9_0123@2 > outL19 ; c out H1.12 < SH1_12_0123@2 > outH112 ; s SL1_9_023@2 1 SL1_9_023@1r
c add H1.3 0123@2 < SH1_3_01@2r SH1_3_23@2 > SH1_3_0123@2 ; s SH1_3_0123@2 3 SH1_3_0123@3r
c add H0.5 023@2 < SH0_5_03@2r PH0_5_2 > SH0_5_023@2 ; c add H0.5 0123@2 < SH0_5_023@2 SH0_5_1@2r > SH0_5_0123@2 ; c out H0.5 < SH0_5_0123@2 > outH05 ; c out H1.3 < SH1_3_0123@2 > outH13 ; s SH0_5_023@2 1 SH0_5_023@1r
c add H0.13 0123@2 < SH0_13_01@2r SH0_13_23@2 > SH0_13_0123@2 ; s SH0_13_0123@2 3 SH0_13_0123@3r
c out L0.1 < SL0_1_0123@2r > outL01 ; c out H0.13 < SH0_13_0123@2 > outH013 ; s SL0_1_0123@2r 1 SL0_1_0123@1r
c add H1.14 0123@2 < SH1_14_01@2r SH1_14_23@2 > SH1_14_0123@2 ; s SH1_14_0123@2 3 SH1_14_0123@3r
c out H1.14 < SH1_14_0123@2 > outH114 ; c out L0.3 < SL0_3_0123@2r > outL03 ; s SL0_3_0123@2r 1 SL0_3_0123@1r
c add L1.0 012@2 < SL1_0_01@2r PL1_0_2 > SL1_0_012@2 ; s SL1_0_012@2 3 SL1_0_012@3r
c add L1.0 0123@2 < SL1_0_012@2 SL1_0_3@2r > SL1_0_0123@2 ; c out L1.0 < SL1_0_0123@2 > outL10 ; c add L1.2 0123@2 < SL1_2_03@2r SL1_2_12@2 > SL1_2_0123@2 ; c out L1.2 < SL1_2_0123@2 > outL12 ; s SL1_2_0123@2 1 SL1_2_0123@1r
c add L1.13 0123@2 < SL1_13_01@2r SL1_13_23@2 > SL1_13_0123@2 ; s SL1_13_0123@2 3 SL1_13_0123@3r
c out L1.13 < SL1_13_0123@2 > outL113 ; c add L1.1 0123@2 < SL1_1_03@2r SL1_1_12@2 > SL1_1_0123@2 ; c out L1.1 < SL1_1_0123@2 > outL11 ; s SL1_1_0123@2 1 SL1_1_0123@1r
c out H0.9 < SH0_9_0123@2r > outH09 ; s SH0_9_0123@2r 3 SH0_9_0123@3r
c add H1.0 0123@2 < SH1_0_03@2r SH1_0_12@2 > SH1_0_0123@2 ; c out H1.0 < SH1_0_0123@2 > outH10 ; s SH1_0_0123@2 1 SH1_0_0123@1r
c add H0.3 012@2 < SH0_3_01@2r PH0_3_2 > SH0_3_012@2 ; s SH0_3_012@2 3 SH0_3_012@3r
c add H1.11 0123@2 < SH1_11_03@2r SH1_11_12@2 > SH1_11_0123@2 ; c out H1.11 < SH1_11_0123@2 > outH111 ; c add H0.3 0123@2 < SH0_3_012@2 SH0_3_3@2r > SH0_3_0123@2 ; c out H0.3 < SH0_3_0123@2 > outH03 ; s SH1_11_0123@2 1 SH1_11_0123@1r
c add H1.2 0123@2 < SH1_2_01@2r SH1_2_23@2 > SH1_2_0123@2 ; s SH1_2_0123@2 3 SH1_2_0123@3r
c out H1.2 < SH1_2_0123@2 > outH12 ; c add H0.1 023@2 < SH0_1_03@2r PH0_1_2 > SH0_1_023@2 ; s SH0_1_023@2 1 SH0_1_023@1r ; c add H0.1 0123@2 < SH0_1_023@2 SH0_1_1@2r > SH0_1_0123@2 ; c out H0.1 < SH0_1_0123@2 > outH01
c add H1.4 012@2 < SH1_4_01@2r PH1_4_2 > SH1_4_012@2 ; s SH1_4_012@2 3 SH1_4_012@3r
c add H1.4 0123@2 < SH1_4_012@2 SH1_4_3@2r > SH1_4_0123@2 ; c out H1.4 < SH1_4_0123@2 > outH14 ; c out H1.8 < SH1_8_0123@2r > outH18
c out H0.4 < SH0_4_0123@2r > outH04 ; s SH0_4_0123@2r 3 SH0_4_0123@3r
c add H1.6 023@2 < SH1_6_03@2r PH1_6_2 > SH1_6_023@2 ; c add H1.6 0123@2 < SH1_6_023@2 SH1_6_1@2r > SH1_6_0123@2 ; c out H1.6 < SH1_6_0123@2 > outH16 ; s SH1_6_023@2 1 SH1_6_023@1r
c out L0.7 < SL0_7_0123@2r > outL07 ; s SL0_7_0123@2r 3 SL0_7_0123@3r
c add H0.0 023@2 < SH0_0_03@2r PH0_0_2 > SH0_0_023@2 ; c add H0.0 0123@2 < SH0_0_023@2 SH0_0_1@2r > SH0_0_0123@2 ; c out H0.0 < SH0_0_0123@2 > outH00 ; s SH0_0_023@2 1 SH0_0_023@1r
c out L1.4 < SL1_4_0123@2r > outL14 ; s SL1_4_0123@2r 3 SL1_4_0123@3r
c add H1.9 0123@2 < SH1_9_03@2r SH1_9_12@2 > SH1_9_0123@2 ; c out H1.9 < SH1_9_0123@2 > outH19 ; s SH1_9_0123@2 1 SH1_9_0123@1r
c add L1.15 0123@2 < SL1_15_01@2r SL1_15_23@2 > SL1_15_0123@2 ; s SL1_15_0123@2 3 SL1_15_0123@3r
c out H1.7 < SH1_7_0123@2r > outH17 ; c out L1.15 < SL1_15_0123@2 > outL115
c out H0.10 < SH0_10_0123@2r > outH010 ; c out L1.7 < SL1_7_0123@2r > outL17
c out H0.2 < SH0_2_0123@2r > outH02 ; c out L0.10 < SL0_10_0123@2r > outL010
c out L1.6 < SL1_6_0123@2r > outL16 ; c out L0.15 < SL0_15_0123@2r > outL015
c out H1.15 < SH1_15_0123@2r > outH115 ; c out H0.14 < SH0_14_0123@2r > outH014
c out L0.2 < SL0_2_0123@2r > outL02 ; c out L0.0 < SL0_0_0123@2r > outL00
c out L1.3 < SL1_3_0123@2r > outL13 ; c out H0.7 < SH0_7_0123@2r > outH07
c out L1.12 < SL1_12_0123@2r > outL112 ; c out H0.12 < SH0_12_0123@2r > outH012
c out H1.5 < SH1_5_0123@2r > outH15 ; c out H0.15 < SH0_15_0123@2r > outH015
c out H0.8 < SH0_8_0123@2r > outH08 ; c out L1.11 < SL1_11_0123@2r > outL111
# chip 3
l raw_wq_a3 ; l raw_wq_a2 ; l raw_wq_a0 ; l raw_x_H0
c cvtq 3a3 < raw_wq_a3 > w3_a3 ; s w3_a3 0 w3_a3
l raw_wq_a1 ; l raw_wq_b ; l raw_x_L0 ; l raw_wo_b1 ; l raw_x_H1 ; c cvtq 3a2 < raw_wq_a2 > w3_a2
l raw_x_L1 ; c cvtq 3a0 < raw_wq_a0 > w3_a0 ; s w3_a0 0 w3_a0
c cvtq 3a1 < raw_wq_a1 > w3_a1
l raw_v_3a0 ; l raw_wo_a0 ; c qproj 3aH0 < raw_x_H0 w3_a0 w3_a1 w3_a2 w3_a3 > q3aH0
s q3aH0 2 q3aH0
l raw_wo_b0 ; l raw_k_0b1 ; c qproj 3bH0 < raw_x_H0 raw_wq_b > q3bH0 ; s w3_a1 0 w3_a1 ; s q3bH0 2 q3bH0
l raw_k_1a0 ; l raw_v_1b0 ; c qproj 3aL0 < raw_x_L0 w3_a0 w3_a1 w3_a2 w3_a3 > q3aL0 ; c qproj 3bL0 < raw_x_L0 raw_wq_b > q3bL0
c cvt wob1 < raw_wo_b1 > wob1
l raw_k_1a1 ; l raw_k_0a1 ; l raw_v_3b0 ; c cq 30 < q3aL0 q3bL0 > cq30 ; s q3bL0 0 q3bL0 ; s cq30 2 cq30
l raw_k_2b0 ; l raw_v_0a1 ; l raw_v_3a1 ; c qproj 3aL1 < raw_x_L1 w3_a0 w3_a1 w3_a2 w3_a3 > q3aL1 ; c qproj 3bH1 < raw_x_H1 raw_wq_b > q3bH1 ; c qproj 3bL1 < raw_x_L1 raw_wq_b > q3bL1
c cvt woa0 < raw_wo_a0 > woa0 ; s q3bH1 2 q3bH1 ; s w3_a2 0 w3_a2
l raw_v_1a1 ; l raw_v_0b1 ; l raw_k_1b0 ; l raw_v_1b1 ; l raw_k_3a0 ; l raw_wo_a1 ; l raw_v_2b0 ; l raw_v_1a0 ; l raw_v_3b1 ; l raw_k_0a0 ; c qproj 3aH1 < raw_x_H1 w3_a0 w3_a1 w3_a2 w3_a3 > q3aH1 ; c cq 31 < q3aL1 q3bL1 > cq31 ; c cvt wob0 < raw_wo_b0 > wob0 ; s q3aH1 2 q3aH1 ; s q3bH0 0 q3bH0 ; s cq31 2 cq31 ; s q3bL1 0 q3bL1
s cq01 2 cq01
l raw_v_2a0 ; l raw_v_2a1 ; c qproj 2bL0 < raw_x_L0 w2_b0 w2_b1 w2_b2 w2_b3 > q2bL0 ; c qproj 2bL1 < raw_x_L1 w2_b0 w2_b1 w2_b2 w2_b3 > q2bL1
l raw_k_1b1 ; s cq00 2 cq00 ; s q2bL1 0 q2bL1
l raw_k_0b0 ; l raw_k_3a1 ; c qproj 2bH0 < raw_x_H0 w2_b0 w2_b1 w2_b2 w2_b3 > q2bH0 ; c att0 2bL0 < q2bL0 k0_2b0_0 k0_2b0_1 v0_2b0_0 v0_2b0_1 > c0_2bL0 ; s c0_2bL0 2 c0_2bL0
s q2aL1 0 q2aL1
l raw_k_2a0 ; l raw_v_0a0 ; c att0 2bH0 < q2bH0 k0_2b0_0 k0_2b0_1 v0_2b0_0 v0_2b0_1 > c0_2bH0
c cvt woa1 < raw_wo_a1 > woa1 ; s c0_2bH0 2 c0_2bH0
l raw_v_0b0 ; l raw_k_2b1 ; l raw_k_2a1 ; c gatt 01 < cq01 raw_k_0a1 raw_k_0b1 raw_v_0a1 raw_v_0b1 > gp01_3
l raw_k_3b0 ; s q2aH1 0 q2aH1 ; s gp01_3 2 gp01_3r
l raw_k_3b1 ; l raw_v_2b1 ; c qproj 2bH1 < raw_x_H1 w2_b0 w2_b1 w2_b2 w2_b3 > q2bH1 ; c gatt 10 < cq10 raw_k_1a0 raw_k_1b0 raw_v_1a0 raw_v_1b0 > gp10_3 ; s q2bH1 0 q2bH1 ; s gp10_3 2 gp10_3r
c gatt 11 < cq11 raw_k_1a1 raw_k_1b1 raw_v_1a1 raw_v_1b1 > gp11_3 ; s gp11_3 2 gp11_3r
c proj 3bL0 < c0_3bL0 wob0 wob1 > ppL0_b ; c cq 21 < q2aL1 q2bL1 > cq21 ; s q3bH1 0 q3bH1
c proj 3aL0 < c0_3aL0 woa0 woa1 > ppL0_a ; c pfin L0 < ppL0_a ppL0_b > PL0_4_3 PL0_5_3 PL0_6_3 PL0_7_3 PL0_8_3 PL0_9_3 PL0_10_3 PL0_11_3 PL0_12_3 PL0_13_3 PL0_14_3 PL0_15_3 ; c add L0.8 03@3 < PL0_8_3 SL0_8_0@3r > SL0_8_03@3 ; c add L0.5 03@3 < PL0_5_3 SL0_5_0@3r > SL0_5_03@3 ; s SL0_5_03@3 2 SL0_5_03@2r
c add L0.14 03@3 < PL0_14_3 SL0_14_0@3r > SL0_14_03@3 ; c add L0.9 03@3 < PL0_9_3 SL0_9_0@3r > SL0_9_03@3 ; c add L0.11 03@3 < PL0_11_3 SL0_11_0@3r > SL0_11_03@3 ; c add L0.12 03@3 < PL0_12_3 SL0_12_0@3r > SL0_12_03@3 ; s PL0_6_3 2 SL0_6_3@2r ; s PL0_13_3 2 SL0_13_3@2r ; s SL0_12_03@3 2 SL0_12_03@2r
c gatt 00 < cq00 raw_k_0a0 raw_k_0b0 raw_v_0a0 raw_v_0b0 > gp00_3 ; c gatt 20 < cq20 raw_k_2a0 raw_k_2b0 raw_v_2a0 raw_v_2b0 > gp20_3 ; s PL0_15_3 0 SL0_15_3@0r ; s PL0_7_3 0 SL0_7_3@0r ; s gp20_3 2 gp20_3r
c zmerge 3bH0 < c0_3bH0 c1_3bH0 > m_3bH0 ; c proj 3bH0 < m_3bH0 wob0 wob1 > ppH0_b
c gmerge 00 < gp00_3 gp00_2r > gacc00_3 ; s gacc00_3 0 gacc00_3r ; s SL0_9_03@3 2 SL0_9_03@2r ; s SL0_8_03@3 2 SL0_8_03@2r
c zmerge 3aH0 < c0_3aH0 c1_3aH0 > m_3aH0 ; c proj 3aH0 < m_3aH0 woa0 woa1 > ppH0_a
c add L0.4 0123@3 < PL0_4_3 SL0_4_0@3r SL0_4_1@3r SL0_4_2@3r > SL0_4_0123@3 ; c out L0.4 < SL0_4_0123@3 > outL04 ; s SL0_4_0123@3 0 SL0_4_0123@0r ; c pfin H0 < ppH0_a ppH0_b > PH0_0_3 PH0_1_3 PH0_2_3 PH0_3_3 PH0_4_3 PH0_5_3 PH0_6_3 PH0_7_3 PH0_8_3 PH0_9_3 PH0_10_3 PH0_11_3 PH0_12_3 PH0_13_3 PH0_14_3 PH0_15_3 ; s PH0_9_3 0 SH0_9_3@0r ; s PH0_4_3 0 SH0_4_3@0r ; s SL0_4_0123@3 2 SL0_4_0123@2r
c add L0.10 23@3 < PL0_10_3 SL0_10_2@3r > SL0_10_23@3 ; s SL0_10_23@3 0 SL0_10_23@0r ; s SL0_11_03@3 2 SL0_11_03@2r
c add H0.10 23@3 < PH0_10_3 SH0_10_2@3r > SH0_10_23@3 ; s SH0_10_23@3 0 SH0_10_23@0r
c add H0.8 23@3 < PH0_8_3 SH0_8_2@3r > SH0_8_23@3 ; s SH0_8_23@3 0 SH0_8_23@0r ; s SL0_14_03@3 2 SL0_14_03@2r
c add H0.12 23@3 < PH0_12_3 SH0_12_2@3r > SH0_12_23@3 ; s SH0_12_23@3 0 SH0_12_23@0r
c add H0.7 23@3 < PH0_7_3 SH0_7_2@3r > SH0_7_23@3 ; s SH0_7_23@3 0 SH0_7_23@0r ; s PH0_13_3 2 SH0_13_3@2r
c add L0.11 123@3 < SL0_11_12@3r PL0_11_3 > SL0_11_123@3 ; c add L0.11 0123@3 < SL0_11_123@3 SL0_11_0@3r > SL0_11_0123@3 ; c out L0.11 < SL0_11_0123@3 > outL011 ; s SL0_11_123@3 0 SL0_11_123@0r
c add H0.2 23@3 < PH0_2_3 SH0_2_2@3r > SH0_2_23@3 ; s SH0_2_23@3 0 SH0_2_23@0r ; s PH0_3_3 2 SH0_3_3@2r
c proj 3aL1 < c0_3aL1 woa0 woa1 > ppL1_a ; c gatt 21 < cq21 raw_k_2a1 raw_k_2b1 raw_v_2a1 raw_v_2b1 > gp21_3
c add L0.5 0123@3 < SL0_5_03@3 SL0_5_12@3r > SL0_5_0123@3 ; c out L0.5 < SL0_5_0123@3 > outL05 ; c add L0.9 0123@3 < SL0_9_03@3 SL0_9_12@3r > SL0_9_0123@3
c add L0.12 0123@3 < SL0_12_03@3 SL0_12_12@3r > SL0_12_0123@3 ; c out L0.9 < SL0_9_0123@3 > outL09 ; c out L0.12 < SL0_12_0123@3 > outL012 ; s SL0_5_0123@3 0 SL0_5_0123@0r ; s SL0_9_0123@3 0 SL0_9_0123@0r ; s SL0_12_0123@3 0 SL0_12_0123@0r ; s gp21_3 2 gp21_3r
c gatt 30 < cq30 raw_k_3a0 raw_k_3b0 raw_v_3a0 raw_v_3b0 > gp30_3 ; c gatt 31 < cq31 raw_k_3a1 raw_k_3b1 raw_v_3a1 raw_v_3b1 > gp31_3
c add L0.8 123@3 < SL0_8_12@3r PL0_8_3 > SL0_8_123@3 ; s SL0_8_123@3 0 SL0_8_123@0r
c add L0.8 0123@3 < SL0_8_123@3 SL0_8_0@3r > SL0_8_0123@3 ; c out L0.8 < SL0_8_0123@3 > outL08 ; c out L0.6 < SL0_6_0123@3r > outL06 ; c add H0.14 23@3 < PH0_14_3 SH0_14_2@3r > SH0_14_23@3 ; s SL0_6_0123@3r 0 SL0_6_0123@0r ; s SH0_14_23@3 0 SH0_14_23@0r ; s PH0_11_3 2 SH0_11_3@2r
c add L0.14 0123@3 < SL0_14_03@3 SL0_14_12@3r > SL0_14_0123@3 ; c out L0.14 < SL0_14_0123@3 > outL014 ; s SL0_14_0123@3 0 SL0_14_0123@0r
c out L0.13 < SL0_13_0123@3r > outL013 ; s SL0_13_0123@3r 0 SL0_13_0123@0r
c proj 3bL1 < c0_3bL1 wob0 wob1 > ppL1_b ; c pfin L1 < ppL1_a ppL1_b > PL1_4_3 PL1_5_3 PL1_6_3 PL1_7_3 PL1_8_3 PL1_9_3 PL1_10_3 PL1_11_3 PL1_12_3 PL1_13_3 PL1_14_3 PL1_15_3 ; s PL1_15_3 2 SL1_15_3@2r ; s PL1_11_3 0 SL1_11_3@0r
c add L1.14 03@3 < PL1_14_3 SL1_14_0@3r > SL1_14_03@3 ; s PL1_8_3 2 SL1_8_3@2r ; s SL1_14_03@3 2 SL1_14_03@2r ; s PL1_4_3 0 SL1_4_3@0r ; s PL1_6_3 2 SL1_6_3@2r ; s PL1_12_3 0 SL1_12_3@0r ; s PL1_5_3 2 SL1_5_3@2r ; s PL1_13_3 2 SL1_13_3@2r
c gfinal 30 < gp30_3 gacc30_2r > gm30 ; c pfing L0 < c0_3aL0 c0_3bL0 gm30 woa0 woa1 wob0 wob1 > PL0_0_3 PL0_1_3 PL0_2_3 PL0_3_3 ; c gfinal 31 < gp31_3 gacc31_2r > gm31 ; c pfing L1 < c0_3aL1 c0_3bL1 gm31 woa0 woa1 wob0 wob1 > PL1_0_3 PL1_1_3 PL1_2_3 PL1_3_3 ; s PL1_0_3 2 SL1_0_3@2r ; s PL1_3_3 2 SL1_3_3@2r ; s PL0_0_3 0 SL0_0_3@0r
c add L0.2 23@3 < PL0_2_3 SL0_2_2@3r > SL0_2_23@3 ; s SL0_2_23@3 0 SL0_2_23@0r
c proj 3bH1 < m_3bH1 wob0 wob1 > ppH1_b
c add H0.5 123@3 < SH0_5_12@3r PH0_5_3 > SH0_5_123@3 ; s SH0_5_123@3 0 SH0_5_123@0r
c add H0.0 123@3 < SH0_0_12@3r PH0_0_3 > SH0_0_123@3 ; s SH0_0_123@3 0 SH0_0_123@0r
c proj 3aH1 < m_3aH1 woa0 woa1 > ppH1_a
c add L1.10 03@3 < PL1_10_3 SL1_10_0@3r > SL1_10_03@3 ; c pfin H1 < ppH1_a ppH1_b > PH1_0_3 PH1_1_3 PH1_2_3 PH1_3_3 PH1_4_3 PH1_5_3 PH1_6_3 PH1_7_3 PH1_8_3 PH1_9_3 PH1_10_3 PH1_11_3 PH1_12_3 PH1_13_3 PH1_14_3 PH1_15_3 ; s PH1_15_3 0 SH1_15_3@0r ; s PH1_14_3 2 SH1_14_3@2r ; s PH1_4_3 2 SH1_4_3@2r ; s PH1_2_3 2 SH1_2_3@2r
c add H0.1 123@3 < SH0_1_12@3r PH0_1_3 > SH0_1_123@3 ; s SH0_1_123@3 0 SH0_1_123@0r
c add H0.6 03@3 < PH0_6_3 SH0_6_0@3r > SH0_6_03@3 ; c add H0.6 0123@3 < SH0_6_03@3 SH0_6_12@3r > SH0_6_0123@3 ; s SH0_6_0123@3 0 SH0_6_0123@0r ; c out H0.6 < SH0_6_0123@3 > outH06 ; s SH0_6_03@3 2 SH0_6_03@2r ; s PH1_12_3 2 SH1_12_3@2r
c add L1.9 123@3 < SL1_9_12@3r PL1_9_3 > SL1_9_123@3 ; s SL1_9_123@3 0 SL1_9_123@0r
c add H0.15 0123@3 < SH0_15_12@3r PH0_15_3 SH0_15_0@3r > SH0_15_0123@3 ; c out H0.15 < SH0_15_0123@3 > outH015 ; s SH0_15_0123@3 0 SH0_15_0123@0r ; s PH1_3_3 2 SH1_3_3@2r
c add L1.7 0123@3 < SL1_7_12@3r PL1_7_3 SL1_7_0@3r > SL1_7_0123@3 ; c out L1.7 < SL1_7_0123@3 > outL17 ; s SL1_7_0123@3 0 SL1_7_0123@0r
c add H0.5 0123@3 < SH0_5_123@3 SH0_5_0@3r > SH0_5_0123@3 ; c out H0.5 < SH0_5_0123@3 > outH05 ; c add H0.5 03@3 < PH0_5_3 SH0_5_0@3r > SH0_5_03@3 ; s SL1_10_03@3 2 SL1_10_03@2r
c add L1.14 123@3 < SL1_14_12@3r PL1_14_3 > SL1_14_123@3 ; c add L1.14 0123@3 < SL1_14_123@3 SL1_14_0@3r > SL1_14_0123@3 ; c out L1.14 < SL1_14_0123@3 > outL114 ; s SL1_14_123@3 0 SL1_14_123@0r
c add L1.9 03@3 < PL1_9_3 SL1_9_0@3r > SL1_9_03@3 ; c add L1.9 0123@3 < SL1_9_123@3 SL1_9_0@3r > SL1_9_0123@3 ; c out L1.9 < SL1_9_0123@3 > outL19 ; s PH1_10_3 2 SH1_10_3@2r
c add L1.10 0123@3 < SL1_10_03@3 SL1_10_12@3r > SL1_10_0123@3 ; c out L1.10 < SL1_10_0123@3 > outL110 ; s SL1_10_0123@3 0 SL1_10_0123@0r
c add H1.13 03@3 < PH1_13_3 SH1_13_0@3r > SH1_13_03@3 ; s SH1_13_03@3 2 SH1_13_03@2r
c add H1.1 03@3 < PH1_1_3 SH1_1_0@3r > SH1_1_03@3 ; s SH1_1_03@3 2 SH1_1_03@2r
c add L0.3 0123@3 < PL0_3_3 SL0_3_0@3r SL0_3_1@3r SL0_3_2@3r > SL0_3_0123@3 ; c out L0.3 < SL0_3_0123@3 > outL03 ; s SL0_3_0123@3 0 SL0_3_0123@0r ; s SL1_9_03@3 2 SL1_9_03@2r
c out L1.8 < SL1_8_0123@3r > outL18 ; s SL1_8_0123@3r 0 SL1_8_0123@0r ; s SH0_5_03@3 2 SH0_5_03@2r
c add L0.1 0123@3 < PL0_1_3 SL0_1_0@3r SL0_1_1@3r SL0_1_2@3r > SL0_1_0123@3 ; c out L0.1 < SL0_1_0123@3 > outL01 ; s SL0_1_0123@3 0 SL0_1_0123@0r ; s SL0_1_0123@3 2 SL0_1_0123@2r
c add H1.5 23@3 < PH1_5_3 SH1_5_2@3r > SH1_5_23@3 ; s SH1_5_23@3 0 SH1_5_23@0r ; s SL0_3_0123@3 2 SL0_3_0123@2r
c add L1.2 03@3 < PL1_2_3 SL1_2_0@3r > SL1_2_03@3 ; c add L1.2 0123@3 < SL1_2_03@3 SL1_2_12@3r > SL1_2_0123@3 ; c out L1.2 < SL1_2_0123@3 > outL12 ; s SL1_2_0123@3 0 SL1_2_0123@0r ; s SL1_2_03@3 2 SL1_2_03@2r
c out L1.5 < SL1_5_0123@3r > outL15 ; s SL1_5_0123@3r 0 SL1_5_0123@0r
c add L1.1 03@3 < PL1_1_3 SL1_1_0@3r > SL1_1_03@3 ; s SL1_1_03@3 2 SL1_1_03@2r
c add H1.0 03@3 < PH1_0_3 SH1_0_0@3r > SH1_0_03@3 ; s SH1_0_03@3 2 SH1_0_03@2r
c add L1.1 0123@3 < SL1_1_03@3 SL1_1_12@3r > SL1_1_0123@3 ; c out L1.1 < SL1_1_0123@3 > outL11 ; s SL1_1_0123@3 0 SL1_1_0123@0r
c add H1.11 03@3 < PH1_11_3 SH1_11_0@3r > SH1_11_03@3 ; s SH1_11_03@3 2 SH1_11_03@2r
c add H1.8 0123@3 < SH1_8_12@3r PH1_8_3 SH1_8_0@3r > SH1_8_0123@3 ; c out H1.8 < SH1_8_0123@3 > outH18 ; s SH1_8_0123@3 0 SH1_8_0123@0r
c add H0.1 0123@3 < SH0_1_123@3 SH0_1_0@3r > SH0_1_0123@3 ; c out H0.1 < SH0_1_0123@3 > outH01 ; c add H0.1 03@3 < PH0_1_3 SH0_1_0@3r > SH0_1_03@3 ; s SH0_1_03@3 2 SH0_1_03@2r
c add H1.6 123@3 < SH1_6_12@3r PH1_6_3 > SH1_6_123@3 ; s SH1_6_123@3 0 SH1_6_123@0r
c out L0.15 < SL0_15_0123@3r > outL015 ; s SH1_8_0123@3 2 SH1_8_0123@2r
c add H1.0 0123@3 < SH1_0_03@3 SH1_0_12@3r > SH1_0_0123@3 ; c out H1.0 < SH1_0_0123@3 > outH10 ; s SH1_0_0123@3 0 SH1_0_0123@0r
c add H1.6 03@3 < PH1_6_3 SH1_6_0@3r > SH1_6_03@3 ; c add H1.6 0123@3 < SH1_6_123@3 SH1_6_0@3r > SH1_6_0123@3 ; c out H1.6 < SH1_6_0123@3 > outH16 ; s SH1_6_03@3 2 SH1_6_03@2r
c add H1.7 0123@3 < SH1_7_12@3r PH1_7_3 SH1_7_0@3r > SH1_7_0123@3 ; c out H1.7 < SH1_7_0123@3 > outH17 ; s SH1_7_0123@3 0 SH1_7_0123@0r
c add H0.0 03@3 < PH0_0_3 SH0_0_0@3r > SH0_0_03@3 ; c add H0.0 0123@3 < SH0_0_123@3 SH0_0_0@3r > SH0_0_0123@3 ; c out H0.0 < SH0_0_0123@3 > outH00 ; s SH0_0_03@3 2 SH0_0_03@2r
c add H1.1 123@3 < SH1_1_12@3r PH1_1_3 > SH1_1_123@3 ; c add H1.1 0123@3 < SH1_1_123@3 SH1_1_0@3r > SH1_1_0123@3 ; s SH1_1_123@3 0 SH1_1_123@0r
c out H1.1 < SH1_1_0123@3 > outH11
c add H1.9 03@3 < PH1_9_3 SH1_9_0@3r > SH1_9_03@3 ; s SH1_9_03@3 2 SH1_9_03@2r
c add H1.9 0123@3 < SH1_9_03@3 SH1_9_12@3r > SH1_9_0123@3 ; c out H1.9 < SH1_9_0123@3 > outH19 ; s SH1_9_0123@3 0 SH1_9_0123@0r
c add H0.12 0123@3 < SH0_12_01@3r SH0_12_23@3 > SH0_12_0123@3 ; c out H0.12 < SH0_12_0123@3 > outH012 ; s SH1_7_0123@3 2 SH1_7_0123@2r
c add H1.11 0123@3 < SH1_11_03@3 SH1_11_12@3r > SH1_11_0123@3 ; c out H1.11 < SH1_11_0123@3 > outH111 ; s SH1_11_0123@3 0 SH1_11_0123@0r
c add H0.14 0123@3 < SH0_14_01@3r SH0_14_23@3 > SH0_14_0123@3 ; c out H0.14 < SH0_14_0123@3 > outH014 ; s SL1_7_0123@3 2 SL1_7_0123@2r
c add H1.13 0123@3 < SH1_13_03@3 SH1_13_12@3r > SH1_13_0123@3 ; s SH1_13_0123@3 0 SH1_13_0123@0r
c out H1.13 < SH1_13_0123@3 > outH113
c add L0.10 0123@3 < SL0_10_01@3r SL0_10_23@3 > SL0_10_0123@3 ; c out L0.10 < SL0_10_0123@3 > outL010 ; s SL0_10_0123@3 2 SL0_10_0123@2r
c out H1.10 < SH1_10_0123@3r > outH110 ; s SH1_10_0123@3r 0 SH1_10_0123@0r
c out H0.2 < SH0_2_0123@3r > outH02 ; s SL0_15_0123@3r 2 SL0_15_0123@2r
c add H0.11 0123@3 < SH0_11_012@3r PH0_11_3 > SH0_11_0123@3 ; c out H0.11 < SH0_11_0123@3 > outH011
c out H0.10 < SH0_10_0123@3r > outH010 ; s SH0_14_0123@3 2 SH0_14_0123@2r
c add H1.12 0123@3 < SH1_12_012@3r PH1_12_3 > SH1_12_0123@3 ; c out H1.12 < SH1_12_0123@3 > outH112
c out L0.0 < SL0_0_0123@3r > outL00 ; s SL0_0_0123@3r 2 SL0_0_0123@2r
c out H1.3 < SH1_3_0123@3r > outH13
c add H0.7 0123@3 < SH0_7_01@3r SH0_7_23@3 > SH0_7_0123@3 ; c out H0.7 < SH0_7_0123@3 > outH07 ; s SH0_7_0123@3 2 SH0_7_0123@2r
c out H0.13 < SH0_13_0123@3r > outH013
c out L0.2 < SL0_2_0123@3r > outL02 ; s SH0_12_0123@3 2 SH0_12_0123@2r
c out H1.14 < SH1_14_0123@3r > outH114
c out H1.5 < SH1_5_0123@3r > outH15 ; s SH0_15_0123@3 2 SH0_15_0123@2r
c add L1.0 0123@3 < SL1_0_012@3r PL1_0_3 > SL1_0_0123@3 ; c out L1.0 < SL1_0_0123@3 > outL10
c out L1.11 < SL1_11_0123@3r > outL111 ; s SL1_11_0123@3r 2 SL1_11_0123@2r
c out L1.13 < SL1_13_0123@3r > outL113
c out H1.15 < SH1_15_0123@3r > outH115
c out H0.9 < SH0_9_0123@3r > outH09
c out L1.6 < SL1_6_0123@3r > outL16
c add H0.3 0123@3 < SH0_3_012@3r PH0_3_3 > SH0_3_0123@3 ; c out H0.3 < SH0_3_0123@3 > outH03
c out H0.8 < SH0_8_0123@3r > outH08
c out H1.2 < SH1_2_0123@3r > outH12
c out L1.12 < SL1_12_0123@3r > outL112
c add H1.4 0123@3 < SH1_4_012@3r PH1_4_3 > SH1_4_0123@3 ; c out H1.4 < SH1_4_0123@3 > outH14
c out L1.3 < SL1_3_0123@3r > outL13
c out H0.4 < SH0_4_0123@3r > outH04
c out L0.7 < SL0_7_0123@3r > outL07
c out L1.4 < SL1_4_0123@3r > outL14
c out L1.15 < SL1_15_0123@3r > outL115
"""


def _parse_prog(text):
    prog, cur = {}, None
    for line in text.strip().split("\n"):
        if line.startswith("# chip"):
            cur = prog.setdefault(int(line.split()[2]), [])
            continue
        step = []
        for op in line.split(" ; "):
            w = op.split()
            if w[0] == "l":
                step.append(("l", w[1]))
            elif w[0] == "s":
                step.append(("s", w[1], int(w[2]), w[3]))
            else:
                i, o = w.index("<"), w.index(">")
                step.append(("c", " ".join(w[1:i]), w[i + 1:o], w[o + 1:]))
        cur.append(step)
    return prog


_KERNEL = make_kernel(_parse_prog(_PROG_TEXT), _NCH, _SPLIT)


def pallas_dist_sparse_attn_localglobal_htp_kvseq_b2_sq256_skv256_hq4_dh64_kernel(x, Wq, K_ext, V_ext, Wo):
    return _KERNEL(x, Wq, K_ext, V_ext, Wo)
```
